```python
import numpy as np

kernel_name = "dist_moe_top2_ep_n2048_d512_e4_h1024"

def setup_inputs():
    x = np.random.randn(2048, 512).astype(np.float32)
    router_W = np.random.randn(512, 16).astype(np.float32) * 0.1
    scores64 = x.astype(np.float64) @ router_W.astype(np.float64)
    route_idx = np.argsort(-scores64, axis=-1)[:, :2].astype(np.int32)
    expert_W = np.random.randn(16, 512, 1024).astype(np.float32) * 0.02
    return {"x": x, "router_W": router_W, "route_idx": route_idx, "expert_W": expert_W}

def reference(x, router_W, route_idx, expert_W):
    scores = x @ router_W
    s_max = scores.max(axis=-1, keepdims=True)
    probs = np.exp(scores - s_max)
    probs = probs / probs.sum(axis=-1, keepdims=True)
    out = np.zeros((2048, 1024), dtype=np.float32)
    for i in range(2048):
        e0, e1 = int(route_idx[i, 0]), int(route_idx[i, 1])
        g0, g1 = probs[i, e0], probs[i, e1]
        gs = g0 + g1
        out[i] = (g0 / gs) * (x[i] @ expert_W[e0]) + (g1 / gs) * (x[i] @ expert_W[e1])
    return out
```

```python
import jax
import jax.numpy as jnp
from jax import lax
from jax.experimental import pallas as pl
from jax.experimental.pallas import tpu as pltpu

N = 2048
D = 512
H = 1024
NCHIP = 4
EL = 4
B = 256
CAP = B // NCHIP
NST = N // B
PRB = B // 64
T = 160
XS_ROWS = 4096 + EL * T
EAGER = 4
MESH = pl.DeviceIdType.MESH


def _iota(shape, d):
    return lax.broadcasted_iota(jnp.int32, shape, d)


def _mm(a, b):
    return jnp.dot(a.astype(jnp.bfloat16), b.astype(jnp.bfloat16),
                   preferred_element_type=jnp.float32)


def _f(m):
    return jnp.where(m, 1.0, 0.0)


def _compress(word, nbits, rows):
    lane = _iota(word.shape, 1)
    for b in range(nbits):
        s = 1 << b
        if s < 128:
            y = pltpu.roll(word, 128 - s, 1)
            y = jnp.where(lane < 128 - s, y, pltpu.roll(y, rows - 1, 0))
        else:
            y = pltpu.roll(word, rows - s // 128, 0)
        word = jnp.where((y & s) != 0, y, jnp.where((word & s) != 0, 0, word))
    return word


def _index_compute(ri, me):
    row = _iota((32, 128), 0)
    lane = _iota((32, 128), 1)
    par = row & 1
    even = par == 0
    chip = ri >> 2
    le = ri & 3
    e0 = jnp.where(even, ri, pltpu.roll(ri, 1, 0))
    e1 = jnp.where(even, pltpu.roll(ri, 31, 0), ri)
    a = e0 >> 2
    b = e1 >> 2
    diff = (b - a) & 3
    nondiag = diff != 2
    pref = jnp.where(diff == 0, a, jnp.where((lane & 1) == 1, a, b))
    r128 = _iota((128, 128), 0)
    c128 = _iota((128, 128), 1)
    uo = jnp.concatenate([_f(r128 < c128), jnp.ones((128, 128), jnp.float32)], axis=1)
    grp = r128 >> 5
    sameg = (r128 >> 5) == (c128 >> 5)
    sameb = (r128 // PRB) == (c128 // PRB)
    lblk = _f(sameb & (c128 < r128))
    bblk = _f(sameb)
    lful = _f(sameg & (c128 < r128))
    bful = _f(sameg)

    def t4(v):
        return jnp.concatenate([v] * 4, axis=0)

    def sel(arr, k):
        return jnp.where(k == 0, arr[0:32], jnp.where(
            k == 1, arr[32:64], jnp.where(k == 2, arr[64:96], arr[96:128])))

    evn4 = (r128 & 1) == 0
    m1 = evn4 & (t4(jnp.where(nondiag, pref, -1)) == grp)
    mem = (t4(chip) == me) & (t4(le) == grp)
    pt = _mm(jnp.concatenate([_f(m1), _f(mem)], axis=0), uo)
    pre1, tot1 = pt[:128, :128], pt[:128, 128:]
    pre_e, tot_e = pt[128:, :128], pt[128:, 128:]
    rank1 = sel((pre1 + _mm(lblk, tot1)).astype(jnp.int32), pref)
    cnt1 = _mm(bblk, tot1).astype(jnp.int32)
    rank_e = (pre_e + _mm(lful, tot_e)).astype(jnp.int32)
    n_e = _mm(bful, tot_e).astype(jnp.int32)
    keep = nondiag & (rank1 < CAP)
    free = CAP - jnp.minimum(cnt1, CAP)
    f1 = free[0:32]
    f2 = f1 + free[32:64]
    f3 = f2 + free[64:96]
    pt2 = _mm(_f(even & jnp.logical_not(keep)), uo)
    rank2 = (pt2[:, :128] + _mm(lblk[:32, :32], pt2[:, 128:])).astype(jnp.int32)
    op = ((rank2 >= f1).astype(jnp.int32) + (rank2 >= f2).astype(jnp.int32)
          + (rank2 >= f3).astype(jnp.int32))
    owner = jnp.where(keep, pref, op)
    owner = jnp.where(even, owner, pltpu.roll(owner, 1, 0))
    pt3 = _mm(_f(evn4 & (t4(owner) == grp)), uo)
    q = sel((pt3[:, :128] + _mm(lblk, pt3[:, 128:])).astype(jnp.int32), owner)
    q = jnp.where(even, q, pltpu.roll(q, 1, 0))
    blk = row // PRB
    v = (blk * (2 * CAP) + par * CAP + q) * 4 + owner
    pos4 = (owner * (N // NCHIP) + blk * CAP + q) * 4
    flat4 = (r128 & 31) * 128 + c128
    word = jnp.where(mem, (flat4 - rank_e) | (t4(v) << 12), 0)
    word = _compress(word, 12, 128)
    valid = flat4 < n_e
    orig = flat4 + (word & 4095)
    lt = jnp.where(valid, ((orig >> 8) * 128 + (orig & 127)) * 4, 0)
    lv = jnp.where(valid, word >> 12, 0)
    flat = row * 128 + lane
    mo = even & (owner == me)
    wo = jnp.where(mo, (flat - (blk * CAP + q)) | (e0 << 12) | (e1 << 16), 0)
    wo = _compress(wo, 12, 32)[:8]
    oo = flat[:8] + (wo & 4095)
    otok4 = jnp.where(row[:8] < 4, ((oo >> 8) * 128 + (oo & 127)) * 4, 0)
    return lt, lv, n_e, pos4, otok4, (wo >> 12) & 15, (wo >> 16) & 15


def _pack(lo, hi):
    ul = lax.bitcast_convert_type(lo, jnp.int32)
    uh = lax.bitcast_convert_type(hi, jnp.int32)
    rl = ul + 0x7FFF + ((ul >> 16) & 1)
    rh = uh + 0x7FFF + ((uh >> 16) & 1)
    return lax.shift_right_logical(rl, 16) | (rh & jnp.int32(-65536))


def _unpack(u):
    lo = lax.bitcast_convert_type(u << 16, jnp.float32)
    hi = lax.bitcast_convert_type(u & jnp.int32(-65536), jnp.float32)
    return lo, hi


def _row(ref, r4):
    return ref.at[pl.ds(pl.multiple_of(r4, 4), 4), :]


def _kernel(x_hbm, rw_hbm, ri_hbm, w_hbm, out_ref,
            xv, xt, wv, riv, rwv, ltv, lvv, posv, otv, oev,
            lts, lvs, poss, ots, cnts,
            xs, pbuf, rbuf, ag, fbuf, xo, g0, g1,
            ld_sems, w_sems, sm_sems, rs_send, rs_recv, ag_send, ag_recv):
    me = lax.axis_index("i")
    left = (me + 3) % NCHIP
    right = (me + 1) % NCHIP

    c_ri = pltpu.make_async_copy(ri_hbm, riv, ld_sems.at[0])
    c_rw = pltpu.make_async_copy(rw_hbm, rwv, ld_sems.at[1])
    c_x = [pltpu.make_async_copy(x_hbm.at[pl.ds(h * 1024, 1024)], xv.at[pl.ds(h * 1024, 1024)],
                                 ld_sems.at[2 + h]) for h in range(2)]
    c_ri.start()

    def start_x(h, c):
        sl = pl.ds(pl.multiple_of(h * 1024, 1024), 1024)
        pltpu.make_async_copy(x_hbm.at[sl], xv.at[sl], ld_sems.at[2 + h]).start()
        return c
    lax.fori_loop(0, 2, start_x, 0)

    def start_w(e, c):
        pltpu.make_async_copy(w_hbm.at[e], wv.at[e], w_sems.at[e]).start(priority=1)
        return c
    lax.fori_loop(0, EL, start_w, 0)
    c_rw.start()

    bar = pltpu.get_barrier_semaphore()
    for k in (1, 2, 3):
        pl.semaphore_signal(bar, inc=1, device_id=((me + k) % NCHIP,), device_id_type=MESH)

    with jax.named_scope("index"):
        c_ri.wait()
        lt, lv, n_e, pos4, otok4, oe0, oe1 = _index_compute(riv[...], me)
        ltv[...] = lt.reshape(128 * 128)
        lvv[...] = lv.reshape(128 * 128)
        posv[...] = pos4.reshape(32 * 128)
        otv[...] = otok4.reshape(8 * 128)
        oev[0:8, :] = oe0
        oev[8:16, :] = oe1
        eager = []
        for e in range(EL):
            sl = pl.ds(e * 4096, EAGER * 128)
            eager.append(pltpu.make_async_copy(ltv.at[sl], lts.at[sl], sm_sems.at[0]))
            eager.append(pltpu.make_async_copy(lvv.at[sl], lvs.at[sl], sm_sems.at[0]))
        eager.append(pltpu.make_async_copy(otv, ots, sm_sems.at[0]))
        for c in eager:
            c.start()
        c_pos = pltpu.make_async_copy(posv, poss, sm_sems.at[1])
        c_pos.start()
        base = jnp.int32(0)
        for e in range(EL):
            n = jnp.max(n_e[e * 32:e * 32 + 8, :])
            cnts[e] = n
            cnts[EL + e] = base
            base = base + ((n + (T - 1)) // T) * T

    for h in range(2):
        with jax.named_scope(f"wait_x{h}"):
            c_x[h].wait()
        with jax.named_scope(f"relayout{h}"):
            for c in range(4):
                xt[pl.ds(h * 4096 + c, 1024, stride=4), :] = xv[h * 1024:(h + 1) * 1024, c * 128:(c + 1) * 128]

    with jax.named_scope("gather"):
        for c in eager:
            c.wait()
        for e in range(EL):
            @pl.when(cnts[e] > EAGER * 128)
            def _(e=e):
                sl = pl.ds(e * 4096 + EAGER * 128, 4096 - EAGER * 128)
                c1 = pltpu.make_async_copy(ltv.at[sl], lts.at[sl], sm_sems.at[2])
                c2 = pltpu.make_async_copy(lvv.at[sl], lvs.at[sl], sm_sems.at[3])
                c1.start()
                c2.start()
                c1.wait()
                c2.wait()

        def gather_e(e, carry):
            n = cnts[e]
            b4 = cnts[EL + e] * 4

            def grp(g, c):
                p0 = g * 16
                l0 = e * 4096 + p0
                vs = [lts[l0 + k] for k in range(16)]
                vals = [xt[pl.ds(pl.multiple_of(vs[k], 4), 4), :] for k in range(16)]
                d0 = pl.multiple_of(b4 + p0 * 4, 64)
                for k in range(16):
                    xs[pl.ds(d0 + k * 4, 4), :] = vals[k]
                return c
            lax.fori_loop(0, (n + 15) >> 4, grp, 0)
            return carry
        lax.fori_loop(0, EL, gather_e, 0)

    with jax.named_scope("gather_owned"):
        def grp_o(g, c):
            p0 = g * 16
            vs = [ots[p0 + k] for k in range(16)]
            vals = [xt[pl.ds(pl.multiple_of(vs[k], 4), 4), :] for k in range(16)]
            d0 = pl.multiple_of(p0 * 4, 64)
            for k in range(16):
                xo[pl.ds(d0 + k * 4, 4), :] = vals[k]
            return c
        lax.fori_loop(0, (N // NCHIP) // 16, grp_o, 0)

    pl.semaphore_wait(bar, 3)

    def rs_copy(src4, v):
        return pltpu.make_async_remote_copy(
            _row(pbuf, src4), _row(rbuf, v & 4092), rs_send, rs_recv.at[v >> 9],
            device_id=v & 3, device_id_type=pl.DeviceIdType.LOGICAL)

    def expert(e, carry):
        n = cnts[e]
        base = cnts[EL + e]
        with jax.named_scope("wait_w"):
            pltpu.make_async_copy(w_hbm.at[e], wv.at[e], w_sems.at[e]).wait()

        def tile(t, c):
            off4 = pl.multiple_of((base + t * T) * 4, 64)
            with jax.named_scope("mm"):
                a = jnp.concatenate(
                    [xs[pl.ds(off4 + cc, T, stride=4), :] for cc in range(4)], axis=1).astype(jnp.bfloat16)
                y = jnp.dot(a, wv[e].astype(jnp.bfloat16), preferred_element_type=jnp.float32)
                pk = _pack(y[:, :512], y[:, 512:])
                for cc in range(4):
                    pbuf[pl.ds(off4 + cc, T, stride=4), :] = pk[:, cc * 128:(cc + 1) * 128]
            with jax.named_scope("rs"):
                nv = jnp.minimum(T, n - t * T)

                def grp(g, c2):
                    l0 = e * 4096 + t * T + g * 8
                    vs = [lvs[l0 + k] for k in range(8)]
                    for k in range(8):
                        rs_copy(off4 + g * 32 + k * 4, vs[k]).start()
                    return c2
                lax.fori_loop(0, nv >> 3, grp, 0)

                def one(k, c2):
                    rs_copy(off4 + k * 4, lvs[e * 4096 + t * T + k]).start()
                    return c2
                lax.fori_loop((nv >> 3) << 3, nv, one, 0)
            return c
        lax.fori_loop(0, (n + (T - 1)) // T, tile, 0)
        return carry
    lax.fori_loop(0, EL, expert, 0)

    with jax.named_scope("router"):
        c_rw.wait()
        rwb = rwv[...].astype(jnp.bfloat16)
        ei = _iota((16, 128), 0)
        w0s, w1s = [], []
        for r in range(4):
            xb = jnp.concatenate(
                [xo[pl.ds(r * 512 + cc, 128, stride=4), :] for cc in range(4)], axis=1).astype(jnp.bfloat16)
            s = lax.dot_general(rwb, xb, (((1,), (1,)), ((), ())), preferred_element_type=jnp.float32)
            p = jnp.exp(s - jnp.max(s, axis=0, keepdims=True))
            probs = p / jnp.sum(p, axis=0, keepdims=True)
            a0 = jnp.sum(jnp.where(ei == oev[r:r + 1, :], probs, 0.0), axis=0, keepdims=True)
            a1 = jnp.sum(jnp.where(ei == oev[8 + r:9 + r, :], probs, 0.0), axis=0, keepdims=True)
            gs = a0 + a1
            w0s.append(a0 / gs)
            w1s.append(a1 / gs)
        wt = jnp.concatenate(w0s + w1s + [jnp.zeros((120, 128), jnp.float32)], axis=0).T
        for r in range(4):
            g0[r * 128:(r + 1) * 128, :] = jnp.broadcast_to(wt[:, r:r + 1], (128, 128))
            g1[r * 128:(r + 1) * 128, :] = jnp.broadcast_to(wt[:, 4 + r:5 + r], (128, 128))

    CH = CAP * 4
    HF = CH // 2

    def chunk(o, j, lo=0, sz=CH):
        return ag.at[pl.ds(pl.multiple_of((o * (N // NCHIP) + j * CAP) * 4 + lo, 8), sz), :]

    def rc(ref, k, dev):
        return pltpu.make_async_remote_copy(ref, ref, ag_send, ag_recv.at[k],
                                            device_id=(dev,), device_id_type=MESH)

    def summ(j):
        with jax.named_scope("wait_r"):
            blk = rbuf.at[pl.ds(j * 2 * CH, 2 * CH), :]
            pltpu.make_async_copy(blk, blk, rs_recv.at[j]).wait()
        with jax.named_scope("sum"):
            ga = g0[j * CAP:(j + 1) * CAP, :]
            gb = g1[j * CAP:(j + 1) * CAP, :]
            dst = pl.multiple_of((me * (N // NCHIP) + j * CAP) * 4, 8)
            for cc in range(4):
                l0, h0 = _unpack(rbuf[pl.ds(j * 2 * CH + cc, CAP, stride=4), :])
                l1, h1 = _unpack(rbuf[pl.ds(j * 2 * CH + CH + cc, CAP, stride=4), :])
                ag[pl.ds(dst + cc, CAP, stride=4), :] = _pack(ga * l0 + gb * l1, ga * h0 + gb * h1)
        rc(chunk(me, j), 4 * j + 0, right).start()
        rc(chunk(me, j), 4 * j + 1, left).start()

    def wait_own(j):
        with jax.named_scope("wait_own"):
            rc(chunk(left, j), 4 * j + 0, right).wait_recv()
            rc(chunk(right, j), 4 * j + 1, left).wait_recv()

    def fwd(j):
        rc(chunk(left, j, 0, HF), 4 * j + 2, right).start()
        rc(chunk(right, j, HF, HF), 4 * j + 3, left).start()

    def finish(j):
        diag = (me + 2) % NCHIP
        with jax.named_scope("wait_fwd"):
            rc(chunk(diag, j, 0, HF), 4 * j + 2, right).wait_recv()
            rc(chunk(diag, j, HF, HF), 4 * j + 3, left).wait_recv()
        with jax.named_scope("unperm"):
            def grp(g, c):
                p0 = g * 16
                l0 = (2 * (j * (B // 128) + (p0 >> 7))) * 128 + (p0 & 127)
                vs = [poss[l0 + k] for k in range(16)]
                vals = [ag[pl.ds(pl.multiple_of(vs[k], 4), 4), :] for k in range(16)]
                d0 = pl.multiple_of(p0 * 4, 64)
                for k in range(16):
                    fbuf[pl.ds(d0 + k * 4, 4), :] = vals[k]
                return c
            lax.fori_loop(0, B // 16, grp, 0)
        with jax.named_scope("unpack"):
            for cc in range(4):
                lo, hi = _unpack(fbuf[pl.ds(cc, B, stride=4), :])
                out_ref[j * B:(j + 1) * B, cc * 128:(cc + 1) * 128] = lo
                out_ref[j * B:(j + 1) * B, 512 + cc * 128:512 + (cc + 1) * 128] = hi

    c_pos.wait()
    summ(0)
    for j in range(NST):
        if j + 1 < NST:
            summ(j + 1)
        wait_own(j)
        fwd(j)
        if j == 0:
            with jax.named_scope("wait_rs_send"):
                ntot = cnts[0] + cnts[1] + cnts[2] + cnts[3]

                def ws16(k, c):
                    blk = pbuf.at[pl.ds(0, 64), :]
                    pltpu.make_async_copy(blk, blk, rs_send).wait()
                    return c
                lax.fori_loop(0, ntot >> 4, ws16, 0)

                def ws(k, c):
                    rs_copy(0, 0).wait_send()
                    return c
                lax.fori_loop(0, ntot & 15, ws, 0)
        if j > 0:
            finish(j - 1)
    finish(NST - 1)

    with jax.named_scope("final"):
        tot = ag.at[pl.ds(0, NST * 3 * CH), :]
        pltpu.make_async_copy(tot, tot, ag_send).wait()


def pallas_dist_moe_top2_ep_n2048_d512_e4_h1024_kernel(x, router_W, route_idx, expert_W):
    rwt = router_W.T
    ri = route_idx.astype(jnp.int32).T.reshape(2, 16, 128).transpose(1, 0, 2).reshape(32, 128)
    i32, f32 = jnp.int32, jnp.float32
    vm, sm = pltpu.VMEM, pltpu.SMEM
    dma = pltpu.SemaphoreType.DMA
    scratch = [
        vm((N, D), f32),
        vm((N * 4, 128), f32),
        vm((EL, D, H), f32),
        vm((32, 128), i32),
        vm((16, D), f32),
        vm((128 * 128,), i32),
        vm((128 * 128,), i32),
        vm((32 * 128,), i32),
        vm((8 * 128,), i32),
        vm((16, 128), i32),
        sm((128 * 128,), i32),
        sm((128 * 128,), i32),
        sm((32 * 128,), i32),
        sm((8 * 128,), i32),
        sm((8,), i32),
        vm((XS_ROWS * 4, 128), f32),
        vm((XS_ROWS * 4, 128), i32),
        vm((1024 * 4, 128), i32),
        vm((N * 4, 128), i32),
        vm((B * 4, 128), i32),
        vm((512 * 4, 128), f32),
        vm((512, 128), f32),
        vm((512, 128), f32),
        dma((4,)), dma((EL,)), dma((4,)), dma, dma((NST,)), dma, dma((4 * NST,)),
    ]
    return pl.pallas_call(
        _kernel,
        out_shape=pltpu.VMEM((N, H), f32),
        in_specs=[pl.BlockSpec(memory_space=pl.ANY)] * 4,
        out_specs=pl.BlockSpec(memory_space=pltpu.VMEM),
        scratch_shapes=scratch,
        compiler_params=pltpu.CompilerParams(collective_id=0, vmem_limit_bytes=100 * 1024 * 1024),
    )(x, rwt, ri, expert_W)
```

```python
import jax
import jax.numpy as jnp
from jax import lax
from jax.experimental import pallas as pl
from jax.experimental.pallas import tpu as pltpu

N = 2048
D = 512
H = 1024
NCHIP = 4
EL = 4
B = 256
CAP = B // NCHIP
NST = N // B
PRB = B // 64
T = 160
NU = 2 * EL
XS_ROWS = 4096 + NU * (T + 16)
SEG = 2048
NSEG = 2 * NU
EAGER = 128
LOGICAL = pl.DeviceIdType.LOGICAL


def _iota(shape, d):
    return lax.broadcasted_iota(jnp.int32, shape, d)


def _mm(a, b):
    return jnp.dot(a.astype(jnp.bfloat16), b.astype(jnp.bfloat16),
                   preferred_element_type=jnp.float32)


def _f(m):
    return jnp.where(m, 1.0, 0.0)


def _compress(word, nbits, rows):
    lane = _iota(word.shape, 1)
    for b in range(nbits):
        s = 1 << b
        if s < 128:
            y = pltpu.roll(word, 128 - s, 1)
            y = jnp.where(lane < 128 - s, y, pltpu.roll(y, rows - 1, 0))
        else:
            y = pltpu.roll(word, rows - s // 128, 0)
        word = jnp.where((y & s) != 0, y, jnp.where((word & s) != 0, 0, word))
    return word


def _index_compute(ri, me):
    row = _iota((32, 128), 0)
    lane = _iota((32, 128), 1)
    par = row & 1
    even = par == 0
    chip = ri >> 2
    le = ri & 3
    e0 = jnp.where(even, ri, pltpu.roll(ri, 1, 0))
    e1 = jnp.where(even, pltpu.roll(ri, 31, 0), ri)
    a = e0 >> 2
    b = e1 >> 2
    diff = (b - a) & 3
    nondiag = diff != 2
    later = (e0 & 3) * 2 + (lane & 1) - (e1 & 3) * 2
    pref = jnp.where(diff == 0, a, jnp.where(later > 0, a, b))
    r128 = _iota((128, 128), 0)
    c128 = _iota((128, 128), 1)
    uo = jnp.concatenate([_f(r128 < c128), jnp.ones((128, 128), jnp.float32)], axis=1)
    grp = r128 >> 5
    sameb = (r128 // PRB) == (c128 // PRB)
    lblk = _f(sameb & (c128 < r128))
    bblk = _f(sameb)

    def tile(v, k):
        return jnp.concatenate([v] * k, axis=0)

    def sel(arr, k):
        return jnp.where(k == 0, arr[0:32], jnp.where(
            k == 1, arr[32:64], jnp.where(k == 2, arr[64:96], arr[96:128])))

    evn4 = (r128 & 1) == 0
    pt = _mm(_f(evn4 & (tile(jnp.where(nondiag, pref, -1), 4) == grp)), uo)
    rank1 = sel((pt[:, :128] + _mm(lblk, pt[:, 128:])).astype(jnp.int32), pref)
    cnt1 = _mm(bblk, pt[:, 128:]).astype(jnp.int32)
    keep = nondiag & (rank1 < CAP)
    free = CAP - jnp.minimum(cnt1, CAP)
    f1 = free[0:32]
    f2 = f1 + free[32:64]
    f3 = f2 + free[64:96]
    pt2 = _mm(_f(even & jnp.logical_not(keep)), uo)
    rank2 = (pt2[:, :128] + _mm(lblk[:32, :32], pt2[:, 128:])).astype(jnp.int32)
    op = ((rank2 >= f1).astype(jnp.int32) + (rank2 >= f2).astype(jnp.int32)
          + (rank2 >= f3).astype(jnp.int32))
    owner = jnp.where(keep, pref, op)
    owner = jnp.where(even, owner, pltpu.roll(owner, 1, 0))
    pt3 = _mm(_f(evn4 & (tile(owner, 4) == grp)), uo)
    q = sel((pt3[:, :128] + _mm(lblk, pt3[:, 128:])).astype(jnp.int32), owner)
    q = jnp.where(even, q, pltpu.roll(q, 1, 0))
    blk = row // PRB
    v = (blk * (2 * CAP) + par * CAP + q) * 4 + owner
    pos4 = (owner * (N // NCHIP) + blk * CAP + q) * 4

    def stack(v):
        return jnp.concatenate([v[0:16], v[0:16], v[16:32], v[16:32]] * EL, axis=0)

    r256 = _iota((256, 128), 0)
    c256 = _iota((256, 128), 1)
    g16 = r256 >> 4
    key = jnp.where(chip == me, le * 2 + (owner == me).astype(jnp.int32), -1)
    mem = stack(key) == (g16 >> 2) * 2 + (g16 & 1)
    pe = _mm(_f(mem), uo)
    rr = _iota((256, 256), 0)
    cc = _iota((256, 256), 1)
    sameg = (rr >> 4) == (cc >> 4)
    rank_e = (pe[:, :128] + _mm(_f(sameg & (cc < rr)), pe[:, 128:])).astype(jnp.int32)
    n_e = _mm(_f(sameg), pe[:, 128:]).astype(jnp.int32)
    flat16 = (r256 & 15) * 128 + c256
    word = jnp.where(mem, (flat16 - rank_e) | (stack(v) << 11), 0)
    word = _compress(word, 11, 256)
    valid = flat16 < n_e
    orig = flat16 + (word & 2047)
    tok = (((g16 >> 1) & 1) * 8 + (orig >> 8)) * 128 + (orig & 127)
    lt = jnp.where(valid, tok * 4, 0)
    lv = jnp.where(valid, word >> 11, 0)

    ro = _iota((32, 256), 0)
    co = _iota((32, 256), 1)
    pick = (((co >> 4) == (ro >> 3) * 4 + ((ro >> 2) & 1) * 2 + 1)
            & ((co & 15) < (ro & 3) * PRB))
    offs = _mm(_f(pick), pe[:, 128:]).astype(jnp.int32)

    flat = row * 128 + lane
    mo = even & (owner == me)
    wo = jnp.where(mo, (flat - (blk * CAP + q)) | (e0 << 12) | (e1 << 16), 0)
    wo = _compress(wo, 12, 32)[:8]
    oo = flat[:8] + (wo & 4095)
    otok4 = jnp.where(row[:8] < 4, ((oo >> 8) * 128 + (oo & 127)) * 4, 0)
    return lt, lv, n_e, jnp.concatenate([pos4, offs], axis=0), otok4, (wo >> 12) & 15, (wo >> 16) & 15


def _pack(lo, hi):
    ul = lax.bitcast_convert_type(lo, jnp.int32)
    uh = lax.bitcast_convert_type(hi, jnp.int32)
    rl = ul + 0x7FFF + ((ul >> 16) & 1)
    rh = uh + 0x7FFF + ((uh >> 16) & 1)
    return lax.shift_right_logical(rl, 16) | (rh & jnp.int32(-65536))


def _unpack(u):
    lo = lax.bitcast_convert_type(u << 16, jnp.float32)
    hi = lax.bitcast_convert_type(u & jnp.int32(-65536), jnp.float32)
    return lo, hi


def _row(ref, r4):
    return ref.at[pl.ds(pl.multiple_of(r4, 4), 4), :]


def _ld(ref, r4):
    return ref[pl.ds(pl.multiple_of(r4, 4), 4), :]


def _move_rows(src, dst, lst, l0, d4, groups):
    def grp(g, c):
        l = l0 + g * 16
        d = d4 + g * 64
        vs = [lst[l + k] for k in range(16)]
        vals = [_ld(src, vs[k]) for k in range(16)]
        for k in range(16):
            dst[pl.ds(pl.multiple_of(d + k * 4, 4), 4), :] = vals[k]
        return c
    lax.fori_loop(0, groups, grp, 0)


def _move_rows_std(src, dst, lst, l0, d0, groups):
    def grp(g, c):
        l = l0 + g * 16
        vs = [lst[l + k] for k in range(16)]
        vals = jnp.concatenate([_ld(src, vs[k]) for k in range(16)], axis=0)
        dst[pl.ds(pl.multiple_of(d0 + g * 16, 16), 16), :] = vals.reshape(16, 512)
        return c
    lax.fori_loop(0, groups, grp, 0)


def _kernel(x_hbm, rw_hbm, ri_hbm, w_hbm, out_ref,
            xv, xt, wv, riv, rwv, ltv, lvv, posv, otv, oev,
            lts, lvs, poss, ots, cnts,
            xs, pbuf, rbuf, ag, fbuf, xo, g0, g1,
            ld_sems, w_sems, sm_sems, rs_send, rs_recv, ag_send, ag_recv):
    me = lax.axis_index("i")
    left = (me + 3) % NCHIP
    right = (me + 1) % NCHIP
    diag = (me + 2) % NCHIP

    c_ri = pltpu.make_async_copy(ri_hbm, riv, ld_sems.at[0])
    c_rw = pltpu.make_async_copy(rw_hbm, rwv, ld_sems.at[1])
    c_ri.start()
    c_rw.start()

    def x_copy(h):
        sl = pl.ds(pl.multiple_of(h * 1024, 1024), 1024)
        return pltpu.make_async_copy(x_hbm.at[sl], xv.at[sl], ld_sems.at[2 + h])

    def w_copy(e):
        return pltpu.make_async_copy(w_hbm.at[e], wv.at[e], w_sems.at[e])

    x_copy(0).start()

    def start_w(e, c):
        w_copy(e).start(priority=1)

        @pl.when(e == 0)
        def _():
            x_copy(1).start(priority=1)
        return c
    lax.fori_loop(0, EL, start_w, 0)

    bar = pltpu.get_barrier_semaphore()
    for k in (1, 2, 3):
        pl.semaphore_signal(bar, inc=1, device_id=(me + k) % NCHIP, device_id_type=LOGICAL)

    with jax.named_scope("index"):
        c_ri.wait()
        lt, lv, n_e, pos4, otok4, oe0, oe1 = _index_compute(riv[...], me)
        ltv[...] = lt.reshape(NSEG * SEG)
        lvv[...] = lv.reshape(NSEG * SEG)
        posv[...] = pos4.reshape(64 * 128)
        otv[...] = otok4.reshape(8 * 128)
        oev[0:8, :] = oe0
        oev[8:16, :] = oe1
        eager = [pltpu.make_async_copy(otv, ots, sm_sems.at[0])]
        for s in range(NSEG):
            sl = pl.ds(s * SEG, EAGER)
            eager.append(pltpu.make_async_copy(ltv.at[sl], lts.at[sl], sm_sems.at[0]))
            eager.append(pltpu.make_async_copy(lvv.at[sl], lvs.at[sl], sm_sems.at[0]))
        for c in eager:
            c.start()
        c_pos = pltpu.make_async_copy(posv, poss, sm_sems.at[1])
        c_pos.start()
        base = jnp.int32(0)
        for u in range(NU):
            nr = jnp.max(n_e[u * 32:u * 32 + 8, :])
            ns = jnp.max(n_e[u * 32 + 16:u * 32 + 24, :])
            cnts[u] = nr
            cnts[NU + u] = ns
            cnts[2 * NU + u] = base
            base = base + ((nr + ns + 15 + (T - 1)) // T) * T

    def relayout(h):
        for c in range(8):
            rows = h * 1024 + c * 128
            xt[pl.ds(rows * 4, 512), :] = xv[pl.ds(rows, 128), :].reshape(512, 128)

    def router(r):
        _move_rows(xt, xo, ots, r * 128, r * 512, 8)
        rwb = rwv[...].astype(jnp.bfloat16)
        ei = _iota((16, 128), 0)
        xb = xo[pl.ds(r * 512, 512), :].reshape(128, D).astype(jnp.bfloat16)
        s = lax.dot_general(rwb, xb, (((1,), (1,)), ((), ())), preferred_element_type=jnp.float32)
        p = jnp.exp(s - jnp.max(s, axis=0, keepdims=True))
        probs = p / jnp.sum(p, axis=0, keepdims=True)
        a0 = jnp.sum(jnp.where(ei == oev[r:r + 1, :], probs, 0.0), axis=0, keepdims=True)
        a1 = jnp.sum(jnp.where(ei == oev[8 + r:9 + r, :], probs, 0.0), axis=0, keepdims=True)
        gs = a0 + a1
        wt = jnp.concatenate([a0 / gs, a1 / gs, jnp.zeros((126, 128), jnp.float32)], axis=0).T
        rows = pl.ds(r * 512, 512)
        g0[rows, :] = jnp.broadcast_to(wt[:, 0:1], (128, 512)).reshape(512, 128)
        g1[rows, :] = jnp.broadcast_to(wt[:, 1:2], (128, 512)).reshape(512, 128)

    def gather_unit(u):
        nr = cnts[u]
        ns = cnts[NU + u]
        b4 = cnts[2 * NU + u] * 4
        _move_rows(xt, xs, lts, u * 2 * SEG, b4, (nr + 15) >> 4)
        _move_rows(xt, xs, lts, (u * 2 + 1) * SEG, b4 + nr * 4, (ns + 15) >> 4)

    with jax.named_scope("wait_x0"):
        x_copy(0).wait()
    with jax.named_scope("relayout0"):
        relayout(0)
    with jax.named_scope("wait_lists"):
        for c in eager:
            c.wait()
        for s in range(NSEG):
            @pl.when(cnts[(s >> 1) + NU * (s & 1)] > EAGER)
            def _(s=s):
                sl = pl.ds(s * SEG + EAGER, SEG - EAGER)
                c1 = pltpu.make_async_copy(ltv.at[sl], lts.at[sl], sm_sems.at[2])
                c2 = pltpu.make_async_copy(lvv.at[sl], lvs.at[sl], sm_sems.at[3])
                c1.start()
                c2.start()
                c1.wait()
                c2.wait()
        c_rw.wait()
    with jax.named_scope("gather0"):
        def gather_e(e, carry):
            gather_unit(2 * e)
            return carry
        lax.fori_loop(0, EL, gather_e, 0)
    pl.semaphore_wait(bar, 3)

    def rs_copy(src4, v):
        return pltpu.make_async_remote_copy(
            _row(pbuf, src4), _row(rbuf, v & 4092), rs_send, rs_recv.at[v >> 9],
            device_id=v & 3, device_id_type=LOGICAL)

    def self_copy(src4, v):
        return pltpu.make_async_copy(_row(pbuf, src4), _row(rbuf, v & 4092), rs_recv.at[v >> 9])

    CH = CAP * 4
    HF = CH // 2

    def chunk(o, j, lo=0, sz=CH):
        return ag.at[pl.ds(pl.multiple_of((o * (N // NCHIP) + j * CAP) * 4 + lo, 8), sz), :]

    def rc(ref, k, dev):
        return pltpu.make_async_remote_copy(ref, ref, ag_send, ag_recv.at[k],
                                            device_id=dev, device_id_type=LOGICAL)

    def self_rows(j):
        def per_expert(e, carry):
            u = 2 * e + j // (NST // 2)
            lo = poss[4096 + (e * 8 + j) * 128]
            hi = poss[4096 + (e * 8 + j + 1) * 128] if (j + 1) % (NST // 2) else cnts[NU + u]
            ls = (u * 2 + 1) * SEG + lo
            s4 = (cnts[2 * NU + u] + cnts[u] + lo) * 4
            cnt = hi - lo

            def sgrp(g, c2):
                vs = [lvs[ls + g * 4 + k] for k in range(4)]
                for k in range(4):
                    self_copy(s4 + g * 16 + k * 4, vs[k]).start()
                return c2
            lax.fori_loop(0, cnt >> 2, sgrp, 0)

            def sone(k, c2):
                self_copy(s4 + k * 4, lvs[ls + k]).start()
                return c2
            lax.fori_loop((cnt >> 2) << 2, cnt, sone, 0)
            return carry
        lax.fori_loop(0, EL, per_expert, 0)

    def summ(j):
        with jax.named_scope("self"):
            self_rows(j)
        with jax.named_scope("wait_r"):
            blk = rbuf.at[pl.ds(j * 2 * CH, 2 * CH), :]
            pltpu.make_async_copy(blk, blk, rs_recv.at[j]).wait()
        with jax.named_scope("sum"):
            ga = g0[j * CH:(j + 1) * CH, :]
            gb = g1[j * CH:(j + 1) * CH, :]
            dst = pl.multiple_of((me * (N // NCHIP) + j * CAP) * 4, 8)
            l0, h0 = _unpack(rbuf[pl.ds(j * 2 * CH, CH), :])
            l1, h1 = _unpack(rbuf[pl.ds(j * 2 * CH + CH, CH), :])
            ag[pl.ds(dst, CH), :] = _pack(ga * l0 + gb * l1, ga * h0 + gb * h1)
        rc(chunk(me, j), 4 * j + 0, right).start()
        rc(chunk(me, j), 4 * j + 1, left).start()

    def wait_own(j):
        with jax.named_scope("wait_own"):
            rc(chunk(left, j), 4 * j + 0, right).wait_recv()
            rc(chunk(right, j), 4 * j + 1, left).wait_recv()

    def fwd(j):
        rc(chunk(left, j, 0, HF), 4 * j + 2, right).start()
        rc(chunk(right, j, HF, HF), 4 * j + 3, left).start()

    def finish(j):
        with jax.named_scope("wait_fwd"):
            rc(chunk(diag, j, 0, HF), 4 * j + 2, right).wait_recv()
            rc(chunk(diag, j, HF, HF), 4 * j + 3, left).wait_recv()
        with jax.named_scope("unperm"):
            for hh in range(B // 128):
                _move_rows_std(ag, fbuf, poss, 2 * (j * (B // 128) + hh) * 128, hh * 128, 8)
        with jax.named_scope("unpack"):
            lo, hi = _unpack(fbuf[...])
            out_ref[j * B:(j + 1) * B, 0:512] = lo
            out_ref[j * B:(j + 1) * B, 512:1024] = hi

    def unit(u, carry):
        e = u >> 1
        nr = cnts[u]
        ns = cnts[NU + u]
        n = nr + ns
        base = cnts[2 * NU + u]

        @pl.when(u == 1)
        def _():
            with jax.named_scope("router"):
                router(0)
            with jax.named_scope("wait_x1"):
                x_copy(1).wait()
            with jax.named_scope("relayout1"):
                relayout(1)

        @pl.when((u & 1) == 1)
        def _():
            with jax.named_scope("gather1"):
                gather_unit(u)

        @pl.when((u & 1) == 0)
        def _():
            with jax.named_scope("wait_w"):
                w_copy(e).wait()

        def tile(t, c):
            p0 = t * T
            off4 = pl.multiple_of((base + p0) * 4, 64)
            with jax.named_scope("mm"):
                a = xs[pl.ds(off4, T * 4), :].reshape(T, D).astype(jnp.bfloat16)
                y = jnp.dot(a, wv[e].astype(jnp.bfloat16), preferred_element_type=jnp.float32)
                pbuf[pl.ds(off4, T * 4), :] = _pack(y[:, :512], y[:, 512:]).reshape(T * 4, 128)
            with jax.named_scope("rs"):
                nrem = jnp.clip(nr - p0, 0, T)
                lr = u * 2 * SEG + p0

                def grp(g, c2):
                    vs = [lvs[lr + g * 8 + k] for k in range(8)]
                    for k in range(8):
                        rs_copy(off4 + g * 32 + k * 4, vs[k]).start()
                    return c2
                lax.fori_loop(0, nrem >> 3, grp, 0)

                def one(k, c2):
                    rs_copy(off4 + k * 4, lvs[lr + k]).start()
                    return c2
                lax.fori_loop((nrem >> 3) << 3, nrem, one, 0)
            return c
        lax.fori_loop(0, (n + (T - 1)) // T, tile, 0)
        return carry
    lax.fori_loop(0, NU, unit, 0)

    c_pos.wait()
    summ(0)
    for j in range(NST):
        if j + 1 < NST:
            summ(j + 1)
        if j < 3:
            with jax.named_scope("router"):
                router(j + 1)
        if j == 0:
            with jax.named_scope("wait_rs_send"):
                ntot = jnp.int32(0)
                for u in range(NU):
                    ntot = ntot + cnts[u]

                def ws16(k, c):
                    blk = pbuf.at[pl.ds(0, 64), :]
                    pltpu.make_async_copy(blk, blk, rs_send).wait()
                    return c
                lax.fori_loop(0, ntot >> 4, ws16, 0)

                def ws(k, c):
                    rs_copy(0, 0).wait_send()
                    return c
                lax.fori_loop(0, ntot & 15, ws, 0)
        wait_own(j)
        fwd(j)
        if j > 0:
            finish(j - 1)
    finish(NST - 1)

    with jax.named_scope("final"):
        tot = ag.at[pl.ds(0, NST * 3 * CH), :]
        pltpu.make_async_copy(tot, tot, ag_send).wait()


def pallas_dist_moe_top2_ep_n2048_d512_e4_h1024_kernel(x, router_W, route_idx, expert_W):
    rwt = router_W.T
    ri = route_idx.astype(jnp.int32).T.reshape(2, 16, 128).transpose(1, 0, 2).reshape(32, 128)
    i32, f32 = jnp.int32, jnp.float32
    vm, sm = pltpu.VMEM, pltpu.SMEM
    dma = pltpu.SemaphoreType.DMA
    scratch = [
        vm((N, D), f32),
        vm((N * 4, 128), f32),
        vm((EL, D, H), f32),
        vm((32, 128), i32),
        vm((16, D), f32),
        vm((NSEG * SEG,), i32),
        vm((NSEG * SEG,), i32),
        vm((64 * 128,), i32),
        vm((8 * 128,), i32),
        vm((16, 128), i32),
        sm((NSEG * SEG,), i32),
        sm((NSEG * SEG,), i32),
        sm((64 * 128,), i32),
        sm((8 * 128,), i32),
        sm((32,), i32),
        vm((XS_ROWS * 4, 128), f32),
        vm((XS_ROWS * 4, 128), i32),
        vm((1024 * 4, 128), i32),
        vm((N * 4, 128), i32),
        vm((B, 512), i32),
        vm((512 * 4, 128), f32),
        vm((512 * 4, 128), f32),
        vm((512 * 4, 128), f32),
        dma((4,)), dma((EL,)), dma((4,)), dma, dma((NST,)), dma, dma((4 * NST,)),
    ]
    return pl.pallas_call(
        _kernel,
        out_shape=pltpu.VMEM((N, H), f32),
        in_specs=[pl.BlockSpec(memory_space=pl.ANY)] * 4,
        out_specs=pl.BlockSpec(memory_space=pltpu.VMEM),
        scratch_shapes=scratch,
        compiler_params=pltpu.CompilerParams(collective_id=0, vmem_limit_bytes=100 * 1024 * 1024,
                                             disable_bounds_checks=True, disable_semaphore_checks=True),
    )(x, rwt, ri, expert_W)
```

```python
import jax
import jax.numpy as jnp
from jax import lax
from jax.experimental import pallas as pl
from jax.experimental.pallas import tpu as pltpu

N = 2048
D = 512
H = 1024
NCHIP = 4
EL = 4
STAGE_ROWS = (1, 1, 2, 2, 2, 2, 2, 2, 1, 1)
NST = len(STAGE_ROWS)
TR0 = tuple(sum(STAGE_ROWS[:j]) for j in range(NST))
CAPS = tuple(32 * r for r in STAGE_ROWS)
PB = tuple(32 * t for t in TR0)
T = 160
NU = 2 * EL
XS_ROWS = 4096 + NU * (T + 16)
SEG = 2048
NSEG = 2 * NU
EAGER = 256
LOGICAL = pl.DeviceIdType.LOGICAL


def _iota(shape, d):
    return lax.broadcasted_iota(jnp.int32, shape, d)


def _mm(a, b):
    return jnp.dot(a.astype(jnp.bfloat16), b.astype(jnp.bfloat16),
                   preferred_element_type=jnp.float32)


def _f(m):
    return jnp.where(m, 1.0, 0.0)


def _by_stage(trow, table):
    out = jnp.full(trow.shape, table[0], jnp.int32)
    for j in range(1, NST):
        if table[j] != table[j - 1]:
            out = out + jnp.where(trow >= TR0[j], table[j] - table[j - 1], 0)
    return out


def _compress(word, nbits, rows):
    lane = _iota(word.shape, 1)
    for b in range(nbits):
        s = 1 << b
        if s < 128:
            y = pltpu.roll(word, 128 - s, 1)
            y = jnp.where(lane < 128 - s, y, pltpu.roll(y, rows - 1, 0))
        else:
            y = pltpu.roll(word, rows - s // 128, 0)
        word = jnp.where((y & s) != 0, y, jnp.where((word & s) != 0, 0, word))
    return word


def _index_compute(ri, me):
    row = _iota((32, 128), 0)
    lane = _iota((32, 128), 1)
    par = row & 1
    even = par == 0
    chip = ri >> 2
    le = ri & 3
    e0 = jnp.where(even, ri, pltpu.roll(ri, 1, 0))
    e1 = jnp.where(even, pltpu.roll(ri, 31, 0), ri)
    a = e0 >> 2
    b = e1 >> 2
    diff = (b - a) & 3
    isdiag = diff == 2
    later = (e0 & 3) * 2 + (lane & 1) - (e1 & 3) * 2
    pref = jnp.where((diff == 0) | (later > 0), a, b)
    other = a + b - pref
    r128 = _iota((128, 128), 0)
    c128 = _iota((128, 128), 1)
    uo = jnp.concatenate([_f(r128 < c128), jnp.ones((128, 128), jnp.float32)], axis=1)
    grp = r128 >> 5
    stages = tuple(range(NST))
    sameb = (((r128 >> 5) == (c128 >> 5))
             & (_by_stage((r128 & 31) >> 1, stages) == _by_stage((c128 & 31) >> 1, stages)))
    cap = _by_stage(row >> 1, CAPS)
    lblk = _f(sameb & (c128 < r128))
    bblk = _f(sameb)

    def tile(v, k):
        return jnp.concatenate([v] * k, axis=0)

    def sel(arr, k):
        return jnp.where(k == 0, arr[0:32], jnp.where(
            k == 1, arr[32:64], jnp.where(k == 2, arr[64:96], arr[96:128])))

    evn4 = (r128 & 1) == 0
    cap4 = tile(cap, 4)

    def ranks(key):
        pt = _mm(_f(evn4 & (tile(key, 4) == grp)), uo)
        rk = (pt[:, :128] + _mm(lblk, pt[:, 128:])).astype(jnp.int32)
        return rk, _mm(bblk, pt[:, 128:]).astype(jnp.int32)

    rk1, cnt1 = ranks(jnp.where(isdiag, -1, pref))
    rk2, cnt2 = ranks(jnp.where(isdiag, pref, -1))
    used1 = jnp.minimum(cnt1, cap4)
    keep = jnp.where(isdiag, sel(rk2 + used1, pref), sel(rk1, pref)) < cap
    free = cap4 - jnp.minimum(cnt1 + cnt2, cap4)
    second = isdiag & jnp.logical_not(keep)
    rk3, cnt3 = ranks(jnp.where(second, other, -1))
    keep2 = second & (sel(rk3 - free, other) < 0)
    free = free - jnp.minimum(cnt3, free)
    f1 = free[0:32]
    f2 = f1 + free[32:64]
    f3 = f2 + free[64:96]
    pt2 = _mm(_f(even & jnp.logical_not(keep | keep2)), uo)
    rank2 = (pt2[:, :128] + _mm(lblk[:32, :32], pt2[:, 128:])).astype(jnp.int32)
    op = ((rank2 >= f1).astype(jnp.int32) + (rank2 >= f2).astype(jnp.int32)
          + (rank2 >= f3).astype(jnp.int32))
    owner = jnp.where(keep, pref, jnp.where(keep2, other, op))
    owner = jnp.where(even, owner, pltpu.roll(owner, 1, 0))
    pt3 = _mm(_f(evn4 & (tile(owner, 4) == grp)), uo)
    q = sel((pt3[:, :128] + _mm(lblk, pt3[:, 128:])).astype(jnp.int32), owner)
    q = jnp.where(even, q, pltpu.roll(q, 1, 0))
    pb = _by_stage(row >> 1, PB)
    v = ((2 * pb + par * cap + q) * 4 + owner) | (_by_stage(row >> 1, stages) << 12)
    pos4 = (owner * (N // NCHIP) + pb + q) * 4

    def stack(v):
        return jnp.concatenate([v[0:16], v[0:16], v[16:32], v[16:32]] * EL, axis=0)

    r256 = _iota((256, 128), 0)
    c256 = _iota((256, 128), 1)
    g16 = r256 >> 4
    key = jnp.where(chip == me, le * 2 + (owner == me).astype(jnp.int32), -1)
    mem = stack(key) == (g16 >> 2) * 2 + (g16 & 1)
    pe = _mm(_f(mem), uo)
    rr = _iota((256, 256), 0)
    cc = _iota((256, 256), 1)
    sameg = (rr >> 4) == (cc >> 4)
    rank_e = (pe[:, :128] + _mm(_f(sameg & (cc < rr)), pe[:, 128:])).astype(jnp.int32)
    n_e = _mm(_f(sameg), pe[:, 128:]).astype(jnp.int32)
    flat16 = (r256 & 15) * 128 + c256
    word = jnp.where(mem, (flat16 - rank_e) | (stack(v) << 11), 0)
    word = _compress(word, 11, 256)
    valid = flat16 < n_e
    orig = flat16 + (word & 2047)
    tok = (((g16 >> 1) & 1) * 8 + (orig >> 8)) * 128 + (orig & 127)
    lt = jnp.where(valid, tok * 4, 0)
    lv = jnp.where(valid, word >> 11, 0)

    ro = _iota((64, 256), 0)
    co = _iota((64, 256), 1)
    jj = ro & 15
    half = jnp.zeros_like(ro)
    start = jnp.zeros_like(ro)
    for j in range(NST):
        half = jnp.where(jj == j, TR0[j] // 8, half)
        start = jnp.where(jj == j, 2 * (TR0[j] % 8), start)
    pick = ((co >> 4) == (ro >> 4) * 4 + half * 2 + 1) & ((co & 15) < start)
    offs = _mm(_f(pick), pe[:, 128:]).astype(jnp.int32)

    flat = row * 128 + lane
    mo = even & (owner == me)
    wo = jnp.where(mo, (flat - (pb + q)) | (e0 << 12) | (e1 << 16), 0)
    wo = _compress(wo, 12, 32)[:8]
    oo = flat[:8] + (wo & 4095)
    otok4 = jnp.where(row[:8] < 4, ((oo >> 8) * 128 + (oo & 127)) * 4, 0)
    return lt, lv, n_e, jnp.concatenate([pos4, offs], axis=0), otok4, (wo >> 12) & 15, (wo >> 16) & 15


def _pack(lo, hi):
    ul = lax.bitcast_convert_type(lo, jnp.int32)
    uh = lax.bitcast_convert_type(hi, jnp.int32)
    rl = ul + 0x7FFF + ((ul >> 16) & 1)
    rh = uh + 0x7FFF + ((uh >> 16) & 1)
    return lax.shift_right_logical(rl, 16) | (rh & jnp.int32(-65536))


def _unpack(u):
    lo = lax.bitcast_convert_type(u << 16, jnp.float32)
    hi = lax.bitcast_convert_type(u & jnp.int32(-65536), jnp.float32)
    return lo, hi


def _row(ref, r4):
    return ref.at[pl.ds(pl.multiple_of(r4, 4), 4), :]


def _ld(ref, r4):
    return ref[pl.ds(pl.multiple_of(r4, 4), 4), :]


def _move_rows(src, dst, lst, l0, d4, groups):
    def grp(g, c):
        l = l0 + g * 16
        d = d4 + g * 64
        vs = [lst[l + k] for k in range(16)]
        vals = [_ld(src, vs[k]) for k in range(16)]
        for k in range(16):
            dst[pl.ds(pl.multiple_of(d + k * 4, 4), 4), :] = vals[k]
        return c
    lax.fori_loop(0, groups, grp, 0)


def _move_rows_std(src, dst, lst, l0, d0, groups):
    def grp(g, c):
        l = l0 + g * 16
        vs = [lst[l + k] for k in range(16)]
        vals = jnp.concatenate([_ld(src, vs[k]) for k in range(16)], axis=0)
        dst[pl.ds(pl.multiple_of(d0 + g * 16, 16), 16), :] = vals.reshape(16, 512)
        return c
    lax.fori_loop(0, groups, grp, 0)


def _kernel(x_hbm, rw_hbm, ri_hbm, w_hbm, out_ref,
            xv, xt, wv, riv, rwv, ltv, lvv, posv, otv, oev,
            lts, lvs, poss, ots, cnts,
            xs, pbuf, rbuf, ag, fbuf, xo, g0, g1,
            ld_sems, w_sems, sm_sems, rs_send, rs_recv, ag_send, ag_recv):
    me = lax.axis_index("i")
    left = (me + 3) % NCHIP
    right = (me + 1) % NCHIP
    diag = (me + 2) % NCHIP

    c_ri = pltpu.make_async_copy(ri_hbm, riv, ld_sems.at[0])
    c_rw = pltpu.make_async_copy(rw_hbm, rwv, ld_sems.at[1])
    c_ri.start()
    c_rw.start()

    def x_copy(h):
        sl = pl.ds(pl.multiple_of(h * 1024, 1024), 1024)
        return pltpu.make_async_copy(x_hbm.at[sl], xv.at[sl], ld_sems.at[2 + h])

    def w_copy(e):
        return pltpu.make_async_copy(w_hbm.at[e], wv.at[e], w_sems.at[e])

    x_copy(0).start()

    def start_w(e, c):
        w_copy(e).start(priority=1)

        @pl.when(e == 0)
        def _():
            x_copy(1).start(priority=1)
        return c
    lax.fori_loop(0, EL, start_w, 0)

    bar = pltpu.get_barrier_semaphore()
    for k in (1, 2, 3):
        pl.semaphore_signal(bar, inc=1, device_id=(me + k) % NCHIP, device_id_type=LOGICAL)

    with jax.named_scope("index"):
        c_ri.wait()
        lt, lv, n_e, pos4, otok4, oe0, oe1 = _index_compute(riv[...], me)
        ltv[...] = lt.reshape(NSEG * SEG)
        lvv[...] = lv.reshape(NSEG * SEG)
        posv[...] = pos4.reshape(96 * 128)
        otv[...] = otok4.reshape(8 * 128)
        oev[0:8, :] = oe0
        oev[8:16, :] = oe1
        eager = [pltpu.make_async_copy(otv, ots, sm_sems.at[0])]
        for s in range(NSEG):
            sl = pl.ds(s * SEG, EAGER)
            eager.append(pltpu.make_async_copy(ltv.at[sl], lts.at[sl], sm_sems.at[0]))
            eager.append(pltpu.make_async_copy(lvv.at[sl], lvs.at[sl], sm_sems.at[0]))
        for c in eager:
            c.start()
        c_pos = pltpu.make_async_copy(posv, poss, sm_sems.at[1])
        c_pos.start()
        base = jnp.int32(0)
        for u in range(NU):
            nr = jnp.max(n_e[u * 32:u * 32 + 8, :])
            ns = jnp.max(n_e[u * 32 + 16:u * 32 + 24, :])
            cnts[u] = nr
            cnts[NU + u] = ns
            cnts[2 * NU + u] = base
            base = base + ((nr + ns + 15 + (T - 1)) // T) * T

    def relayout(h):
        for c in range(8):
            rows = h * 1024 + c * 128
            xt[pl.ds(rows * 4, 512), :] = xv[pl.ds(rows, 128), :].reshape(512, 128)

    def router(r):
        _move_rows(xt, xo, ots, r * 128, r * 512, 8)
        rwb = rwv[...].astype(jnp.bfloat16)
        ei = _iota((16, 128), 0)
        xb = xo[pl.ds(r * 512, 512), :].reshape(128, D).astype(jnp.bfloat16)
        s = lax.dot_general(rwb, xb, (((1,), (1,)), ((), ())), preferred_element_type=jnp.float32)
        p = jnp.exp(s - jnp.max(s, axis=0, keepdims=True))
        probs = p / jnp.sum(p, axis=0, keepdims=True)
        a0 = jnp.sum(jnp.where(ei == oev[r:r + 1, :], probs, 0.0), axis=0, keepdims=True)
        a1 = jnp.sum(jnp.where(ei == oev[8 + r:9 + r, :], probs, 0.0), axis=0, keepdims=True)
        gs = a0 + a1
        wt = jnp.concatenate([a0 / gs, a1 / gs, jnp.zeros((126, 128), jnp.float32)], axis=0).T
        rows = pl.ds(r * 512, 512)
        g0[rows, :] = jnp.broadcast_to(wt[:, 0:1], (128, 512)).reshape(512, 128)
        g1[rows, :] = jnp.broadcast_to(wt[:, 1:2], (128, 512)).reshape(512, 128)

    def gather_unit(u):
        nr = cnts[u]
        ns = cnts[NU + u]
        b4 = cnts[2 * NU + u] * 4
        _move_rows(xt, xs, lts, u * 2 * SEG, b4, (nr + 15) >> 4)
        _move_rows(xt, xs, lts, (u * 2 + 1) * SEG, b4 + nr * 4, (ns + 15) >> 4)

    with jax.named_scope("wait_x0"):
        x_copy(0).wait()
    with jax.named_scope("relayout0"):
        relayout(0)
    with jax.named_scope("wait_lists"):
        for c in eager:
            c.wait()
        for s in range(NSEG):
            @pl.when(cnts[(s >> 1) + NU * (s & 1)] > EAGER)
            def _(s=s):
                sl = pl.ds(s * SEG + EAGER, SEG - EAGER)
                c1 = pltpu.make_async_copy(ltv.at[sl], lts.at[sl], sm_sems.at[2])
                c2 = pltpu.make_async_copy(lvv.at[sl], lvs.at[sl], sm_sems.at[3])
                c1.start()
                c2.start()
                c1.wait()
                c2.wait()
        c_rw.wait()
    with jax.named_scope("gather0"):
        def gather_e(e, carry):
            gather_unit(2 * e)
            return carry
        lax.fori_loop(0, EL, gather_e, 0)
    pl.semaphore_wait(bar, 3)

    def rs_copy(src4, v):
        return pltpu.make_async_remote_copy(
            _row(pbuf, src4), _row(rbuf, v & 4092), rs_send, rs_recv.at[v >> 12],
            device_id=v & 3, device_id_type=LOGICAL)

    def self_copy(src4, v):
        return pltpu.make_async_copy(_row(pbuf, src4), _row(rbuf, v & 4092), rs_recv.at[v >> 12])

    def chunk(o, j, part=None):
        sz = CAPS[j] * 4 if part is None else CAPS[j] * 2
        lo = 0 if part is None else part * sz
        return ag.at[pl.ds(pl.multiple_of((o * (N // NCHIP) + PB[j]) * 4 + lo, 8), sz), :]

    def rc(ref, k, dev):
        return pltpu.make_async_remote_copy(ref, ref, ag_send, ag_recv.at[k],
                                            device_id=dev, device_id_type=LOGICAL)

    def self_rows(j):
        h = TR0[j] // 8
        last_in_half = j + 1 == NST or TR0[j + 1] // 8 != h

        def per_expert(e, carry):
            u = 2 * e + h
            lo = poss[4096 + (e * 16 + j) * 128]
            hi = cnts[NU + u] if last_in_half else poss[4096 + (e * 16 + j + 1) * 128]
            ls = (u * 2 + 1) * SEG + lo
            s4 = (cnts[2 * NU + u] + cnts[u] + lo) * 4
            cnt = hi - lo

            def sgrp(g, c2):
                vs = [lvs[ls + g * 4 + k] for k in range(4)]
                for k in range(4):
                    self_copy(s4 + g * 16 + k * 4, vs[k]).start()
                return c2
            lax.fori_loop(0, cnt >> 2, sgrp, 0)

            def sone(k, c2):
                self_copy(s4 + k * 4, lvs[ls + k]).start()
                return c2
            lax.fori_loop((cnt >> 2) << 2, cnt, sone, 0)
            return carry
        lax.fori_loop(0, EL, per_expert, 0)

    def summ(j):
        ch = CAPS[j] * 4
        r0 = PB[j] * 8
        with jax.named_scope("self"):
            self_rows(j)
        with jax.named_scope("wait_r"):
            blk = rbuf.at[pl.ds(r0, 2 * ch), :]
            pltpu.make_async_copy(blk, blk, rs_recv.at[j]).wait()
        with jax.named_scope("sum"):
            ga = g0[PB[j] * 4:PB[j] * 4 + ch, :]
            gb = g1[PB[j] * 4:PB[j] * 4 + ch, :]
            dst = pl.multiple_of((me * (N // NCHIP) + PB[j]) * 4, 8)
            l0, h0 = _unpack(rbuf[pl.ds(r0, ch), :])
            l1, h1 = _unpack(rbuf[pl.ds(r0 + ch, ch), :])
            ag[pl.ds(dst, ch), :] = _pack(ga * l0 + gb * l1, ga * h0 + gb * h1)
        rc(chunk(me, j), 4 * j + 0, right).start()
        rc(chunk(me, j), 4 * j + 1, left).start()

    def wait_own(j):
        with jax.named_scope("wait_own"):
            rc(chunk(left, j), 4 * j + 0, right).wait_recv()
            rc(chunk(right, j), 4 * j + 1, left).wait_recv()

    def fwd(j):
        rc(chunk(left, j, 0), 4 * j + 2, right).start()
        rc(chunk(right, j, 1), 4 * j + 3, left).start()

    def finish(j):
        ntok = STAGE_ROWS[j] * 128
        with jax.named_scope("wait_fwd"):
            rc(chunk(diag, j, 0), 4 * j + 2, right).wait_recv()
            rc(chunk(diag, j, 1), 4 * j + 3, left).wait_recv()
        with jax.named_scope("unperm"):
            for hh in range(STAGE_ROWS[j]):
                _move_rows_std(ag, fbuf, poss, 2 * (TR0[j] + hh) * 128, hh * 128, 8)
        with jax.named_scope("unpack"):
            lo, hi = _unpack(fbuf[0:ntok, :])
            out_ref[TR0[j] * 128:TR0[j] * 128 + ntok, 0:512] = lo
            out_ref[TR0[j] * 128:TR0[j] * 128 + ntok, 512:1024] = hi

    def unit(u, carry):
        e = u >> 1
        nr = cnts[u]
        ns = cnts[NU + u]
        n = nr + ns
        base = cnts[2 * NU + u]

        @pl.when(u == 1)
        def _():
            with jax.named_scope("router"):
                router(0)
            with jax.named_scope("wait_x1"):
                x_copy(1).wait()
            with jax.named_scope("relayout1"):
                relayout(1)

        @pl.when((u & 1) == 1)
        def _():
            with jax.named_scope("gather1"):
                gather_unit(u)

        @pl.when((u & 1) == 0)
        def _():
            with jax.named_scope("wait_w"):
                w_copy(e).wait()

        def tile(t, c):
            p0 = t * T
            off4 = pl.multiple_of((base + p0) * 4, 64)
            with jax.named_scope("mm"):
                a = xs[pl.ds(off4, T * 4), :].reshape(T, D).astype(jnp.bfloat16)
                y = jnp.dot(a, wv[e].astype(jnp.bfloat16), preferred_element_type=jnp.float32)
                pbuf[pl.ds(off4, T * 4), :] = _pack(y[:, :512], y[:, 512:]).reshape(T * 4, 128)
            with jax.named_scope("rs"):
                nrem = jnp.clip(nr - p0, 0, T)
                lr = u * 2 * SEG + p0

                def grp(g, c2):
                    vs = [lvs[lr + g * 8 + k] for k in range(8)]
                    for k in range(8):
                        rs_copy(off4 + g * 32 + k * 4, vs[k]).start()
                    return c2
                lax.fori_loop(0, nrem >> 3, grp, 0)

                def one(k, c2):
                    rs_copy(off4 + k * 4, lvs[lr + k]).start()
                    return c2
                lax.fori_loop((nrem >> 3) << 3, nrem, one, 0)
            return c
        lax.fori_loop(0, (n + (T - 1)) // T, tile, 0)
        return carry
    lax.fori_loop(0, NU, unit, 0)

    c_pos.wait()
    summ(0)
    summ(1)
    next_router = 1
    for j in range(NST):
        if j + 2 < NST:
            summ(j + 2)
        if j + 3 < NST and PB[j + 3] + CAPS[j + 3] > 128 * next_router:
            with jax.named_scope("router"):
                router(next_router)
            next_router += 1
        if j == 0:
            with jax.named_scope("wait_rs_send"):
                ntot = jnp.int32(0)
                for u in range(NU):
                    ntot = ntot + cnts[u]

                def ws16(k, c):
                    blk = pbuf.at[pl.ds(0, 64), :]
                    pltpu.make_async_copy(blk, blk, rs_send).wait()
                    return c
                lax.fori_loop(0, ntot >> 4, ws16, 0)

                def ws(k, c):
                    rs_copy(0, 0).wait_send()
                    return c
                lax.fori_loop(0, ntot & 15, ws, 0)
        wait_own(j)
        fwd(j)
        if 0 < j < NST - 2:
            finish(j - 1)
    finish(NST - 3)
    finish(NST - 2)
    finish(NST - 1)

    with jax.named_scope("final"):
        tot = ag.at[pl.ds(0, 3 * (N // NCHIP) * 4), :]
        pltpu.make_async_copy(tot, tot, ag_send).wait()


def pallas_dist_moe_top2_ep_n2048_d512_e4_h1024_kernel(x, router_W, route_idx, expert_W):
    rwt = router_W.T
    ri = route_idx.astype(jnp.int32).T.reshape(2, 16, 128).transpose(1, 0, 2).reshape(32, 128)
    i32, f32 = jnp.int32, jnp.float32
    vm, sm = pltpu.VMEM, pltpu.SMEM
    dma = pltpu.SemaphoreType.DMA
    scratch = [
        vm((N, D), f32),
        vm((N * 4, 128), f32),
        vm((EL, D, H), f32),
        vm((32, 128), i32),
        vm((16, D), f32),
        vm((NSEG * SEG,), i32),
        vm((NSEG * SEG,), i32),
        vm((96 * 128,), i32),
        vm((8 * 128,), i32),
        vm((16, 128), i32),
        sm((NSEG * SEG,), i32),
        sm((NSEG * SEG,), i32),
        sm((96 * 128,), i32),
        sm((8 * 128,), i32),
        sm((32,), i32),
        vm((XS_ROWS * 4, 128), f32),
        vm((XS_ROWS * 4, 128), i32),
        vm((1024 * 4, 128), i32),
        vm((N * 4, 128), i32),
        vm((256, 512), i32),
        vm((512 * 4, 128), f32),
        vm((512 * 4, 128), f32),
        vm((512 * 4, 128), f32),
        dma((4,)), dma((EL,)), dma((4,)), dma, dma((NST,)), dma, dma((4 * NST,)),
    ]
    return pl.pallas_call(
        _kernel,
        out_shape=pltpu.VMEM((N, H), f32),
        in_specs=[pl.BlockSpec(memory_space=pl.ANY)] * 4,
        out_specs=pl.BlockSpec(memory_space=pltpu.VMEM),
        scratch_shapes=scratch,
        compiler_params=pltpu.CompilerParams(collective_id=0, vmem_limit_bytes=100 * 1024 * 1024,
                                             disable_bounds_checks=True, disable_semaphore_checks=True),
    )(x, rwt, ri, expert_W)
```

```python
import jax
import jax.numpy as jnp
from jax import lax
from jax.experimental import pallas as pl
from jax.experimental.pallas import tpu as pltpu

N = 2048
D = 512
H = 1024
NCHIP = 4
EL = 4
STAGE_ROWS = (1, 1, 2, 2, 2, 2, 2, 2, 1, 1)
NST = len(STAGE_ROWS)
TR0 = tuple(sum(STAGE_ROWS[:j]) for j in range(NST))
CAPS = tuple(32 * r for r in STAGE_ROWS)
PB = tuple(32 * t for t in TR0)
T = 160
NU = 2 * EL
XS_ROWS = 4096 + NU * (T + 16)
SEG = 2048
NSEG = 2 * NU
EAGER = 256
LOGICAL = pl.DeviceIdType.LOGICAL


def _iota(shape, d):
    return lax.broadcasted_iota(jnp.int32, shape, d)


def _mm(a, b):
    return jnp.dot(a.astype(jnp.bfloat16), b.astype(jnp.bfloat16),
                   preferred_element_type=jnp.float32)


def _f(m):
    return jnp.where(m, 1.0, 0.0)


def _by_stage(trow, table):
    out = jnp.full(trow.shape, table[0], jnp.int32)
    for j in range(1, NST):
        if table[j] != table[j - 1]:
            out = out + jnp.where(trow >= TR0[j], table[j] - table[j - 1], 0)
    return out


def _compress(word, nbits, rows):
    lane = _iota(word.shape, 1)
    for b in range(nbits):
        s = 1 << b
        if s < 128:
            y = pltpu.roll(word, 128 - s, 1)
            y = jnp.where(lane < 128 - s, y, pltpu.roll(y, rows - 1, 0))
        else:
            y = pltpu.roll(word, rows - s // 128, 0)
        word = jnp.where((y & s) != 0, y, jnp.where((word & s) != 0, 0, word))
    return word


def _index_compute(ri, me):
    row = _iota((32, 128), 0)
    lane = _iota((32, 128), 1)
    par = row & 1
    even = par == 0
    chip = ri >> 2
    le = ri & 3
    e0 = jnp.where(even, ri, pltpu.roll(ri, 1, 0))
    e1 = jnp.where(even, pltpu.roll(ri, 31, 0), ri)
    a = e0 >> 2
    b = e1 >> 2
    diff = (b - a) & 3
    isdiag = diff == 2
    later = (e0 & 3) * 2 + (lane & 1) - (e1 & 3) * 2
    pref = jnp.where((diff == 0) | (later > 0), a, b)
    other = a + b - pref
    r128 = _iota((128, 128), 0)
    c128 = _iota((128, 128), 1)
    uo = jnp.concatenate([_f(r128 < c128), jnp.ones((128, 128), jnp.float32)], axis=1)
    grp = r128 >> 5
    stages = tuple(range(NST))
    sameb = (((r128 >> 5) == (c128 >> 5))
             & (_by_stage((r128 & 31) >> 1, stages) == _by_stage((c128 & 31) >> 1, stages)))
    cap = _by_stage(row >> 1, CAPS)
    lblk = _f(sameb & (c128 < r128))
    bblk = _f(sameb)

    def tile(v, k):
        return jnp.concatenate([v] * k, axis=0)

    def sel(arr, k):
        return jnp.where(k == 0, arr[0:32], jnp.where(
            k == 1, arr[32:64], jnp.where(k == 2, arr[64:96], arr[96:128])))

    evn4 = (r128 & 1) == 0
    cap4 = tile(cap, 4)

    def ranks(key):
        pt = _mm(_f(evn4 & (tile(key, 4) == grp)), uo)
        rk = (pt[:, :128] + _mm(lblk, pt[:, 128:])).astype(jnp.int32)
        return rk, _mm(bblk, pt[:, 128:]).astype(jnp.int32)

    rk1, cnt1 = ranks(jnp.where(isdiag, -1, pref))
    rk2, cnt2 = ranks(jnp.where(isdiag, pref, -1))
    used1 = jnp.minimum(cnt1, cap4)
    keep = jnp.where(isdiag, sel(rk2 + used1, pref), sel(rk1, pref)) < cap
    free = cap4 - jnp.minimum(cnt1 + cnt2, cap4)
    second = isdiag & jnp.logical_not(keep)
    rk3, cnt3 = ranks(jnp.where(second, other, -1))
    keep2 = second & (sel(rk3 - free, other) < 0)
    free = free - jnp.minimum(cnt3, free)
    f1 = free[0:32]
    f2 = f1 + free[32:64]
    f3 = f2 + free[64:96]
    pt2 = _mm(_f(even & jnp.logical_not(keep | keep2)), uo)
    rank2 = (pt2[:, :128] + _mm(lblk[:32, :32], pt2[:, 128:])).astype(jnp.int32)
    op = ((rank2 >= f1).astype(jnp.int32) + (rank2 >= f2).astype(jnp.int32)
          + (rank2 >= f3).astype(jnp.int32))
    owner = jnp.where(keep, pref, jnp.where(keep2, other, op))
    owner = jnp.where(even, owner, pltpu.roll(owner, 1, 0))
    pt3 = _mm(_f(evn4 & (tile(owner, 4) == grp)), uo)
    q = sel((pt3[:, :128] + _mm(lblk, pt3[:, 128:])).astype(jnp.int32), owner)
    q = jnp.where(even, q, pltpu.roll(q, 1, 0))
    pb = _by_stage(row >> 1, PB)
    v = ((2 * pb + par * cap + q) * 4 + owner) | (_by_stage(row >> 1, stages) << 12)
    pos4 = (owner * (N // NCHIP) + pb + q) * 4

    def stack(v):
        return jnp.concatenate([v[0:16], v[0:16], v[16:32], v[16:32]] * EL, axis=0)

    r256 = _iota((256, 128), 0)
    c256 = _iota((256, 128), 1)
    g16 = r256 >> 4
    key = jnp.where(chip == me, le * 2 + (owner == me).astype(jnp.int32), -1)
    mem = stack(key) == (g16 >> 2) * 2 + (g16 & 1)
    pe = _mm(_f(mem), uo)
    rr = _iota((256, 256), 0)
    cc = _iota((256, 256), 1)
    sameg = (rr >> 4) == (cc >> 4)
    rank_e = (pe[:, :128] + _mm(_f(sameg & (cc < rr)), pe[:, 128:])).astype(jnp.int32)
    n_e = _mm(_f(sameg), pe[:, 128:]).astype(jnp.int32)
    flat16 = (r256 & 15) * 128 + c256
    word = jnp.where(mem, (flat16 - rank_e) | (stack(v) << 11), 0)
    word = _compress(word, 11, 256)
    valid = flat16 < n_e
    orig = flat16 + (word & 2047)
    tok = (((g16 >> 1) & 1) * 8 + (orig >> 8)) * 128 + (orig & 127)
    lt = jnp.where(valid, tok * 4, 0)
    lv = jnp.where(valid, word >> 11, 0)

    ro = _iota((64, 256), 0)
    co = _iota((64, 256), 1)
    jj = ro & 15
    half = jnp.zeros_like(ro)
    start = jnp.zeros_like(ro)
    for j in range(NST):
        half = jnp.where(jj == j, TR0[j] // 8, half)
        start = jnp.where(jj == j, 2 * (TR0[j] % 8), start)
    pick = ((co >> 4) == (ro >> 4) * 4 + half * 2 + 1) & ((co & 15) < start)
    offs = _mm(_f(pick), pe[:, 128:]).astype(jnp.int32)

    flat = row * 128 + lane
    mo = even & (owner == me)
    wo = jnp.where(mo, (flat - (pb + q)) | (e0 << 12) | (e1 << 16), 0)
    wo = _compress(wo, 12, 32)[:8]
    oo = flat[:8] + (wo & 4095)
    otok4 = jnp.where(row[:8] < 4, ((oo >> 8) * 128 + (oo & 127)) * 4, 0)
    return lt, lv, n_e, jnp.concatenate([pos4, offs], axis=0), otok4, (wo >> 12) & 15, (wo >> 16) & 15


def _pack(lo, hi):
    ul = lax.bitcast_convert_type(lo, jnp.int32)
    uh = lax.bitcast_convert_type(hi, jnp.int32)
    rl = ul + 0x7FFF + ((ul >> 16) & 1)
    rh = uh + 0x7FFF + ((uh >> 16) & 1)
    return lax.shift_right_logical(rl, 16) | (rh & jnp.int32(-65536))


def _unpack(u):
    lo = lax.bitcast_convert_type(u << 16, jnp.float32)
    hi = lax.bitcast_convert_type(u & jnp.int32(-65536), jnp.float32)
    return lo, hi


def _row(ref, r4):
    return ref.at[pl.ds(pl.multiple_of(r4, 4), 4), :]


def _ld(ref, r4):
    return ref[pl.ds(pl.multiple_of(r4, 4), 4), :]


def _move_rows(src, dst, lst, l0, d4, groups):
    def grp(g, c):
        l = l0 + g * 16
        d = d4 + g * 64
        vs = [lst[l + k] for k in range(16)]
        vals = [_ld(src, vs[k]) for k in range(16)]
        for k in range(16):
            dst[pl.ds(pl.multiple_of(d + k * 4, 4), 4), :] = vals[k]
        return c
    lax.fori_loop(0, groups, grp, 0)


def _move_rows_std(src, dst, lst, l0, d0, groups):
    def grp(g, c):
        l = l0 + g * 16
        vs = [lst[l + k] for k in range(16)]
        vals = jnp.concatenate([_ld(src, vs[k]) for k in range(16)], axis=0)
        dst[pl.ds(pl.multiple_of(d0 + g * 16, 16), 16), :] = vals.reshape(16, 512)
        return c
    lax.fori_loop(0, groups, grp, 0)


def _kernel(x_hbm, rw_hbm, ri_hbm, w_hbm, out_ref,
            xv, xt, wv, riv, rwv, ltv, lvv, posv, otv, oev,
            lts, lvs, poss, ots, cnts,
            xs, pbuf, rbuf, ag, fbuf, xo, g0, g1,
            ld_sems, w_sems, sm_sems, rs_send, rs_recv, ag_send, ag_recv):
    me = lax.axis_index("i")
    left = (me + 3) % NCHIP
    right = (me + 1) % NCHIP
    diag = (me + 2) % NCHIP

    c_ri = pltpu.make_async_copy(ri_hbm, riv, ld_sems.at[0])
    c_rw = pltpu.make_async_copy(rw_hbm, rwv, ld_sems.at[1])
    c_ri.start()
    c_rw.start()

    def x_copy(h):
        sl = pl.ds(pl.multiple_of(h * 1024, 1024), 1024)
        return pltpu.make_async_copy(x_hbm.at[sl], xv.at[sl], ld_sems.at[2 + h])

    def w_copy(e):
        return pltpu.make_async_copy(w_hbm.at[e], wv.at[e], w_sems.at[e])

    x_copy(0).start()

    def start_w(e, c):
        w_copy(e).start(priority=1)

        @pl.when(e == 0)
        def _():
            x_copy(1).start(priority=1)
        return c
    lax.fori_loop(0, EL, start_w, 0)

    bar = pltpu.get_barrier_semaphore()
    for k in (1, 2, 3):
        pl.semaphore_signal(bar, inc=1, device_id=(me + k) % NCHIP, device_id_type=LOGICAL)

    c_ri.wait()
    lt, lv, n_e, pos4, otok4, oe0, oe1 = _index_compute(riv[...], me)
    ltv[...] = lt.reshape(NSEG * SEG)
    lvv[...] = lv.reshape(NSEG * SEG)
    posv[...] = pos4.reshape(96 * 128)
    otv[...] = otok4.reshape(8 * 128)
    oev[0:8, :] = oe0
    oev[8:16, :] = oe1
    eager = [pltpu.make_async_copy(otv, ots, sm_sems.at[0])]
    for s in range(NSEG):
        sl = pl.ds(s * SEG, EAGER)
        eager.append(pltpu.make_async_copy(ltv.at[sl], lts.at[sl], sm_sems.at[0]))
        eager.append(pltpu.make_async_copy(lvv.at[sl], lvs.at[sl], sm_sems.at[0]))
    for c in eager:
        c.start()
    c_pos = pltpu.make_async_copy(posv, poss, sm_sems.at[1])
    c_pos.start()
    base = jnp.int32(0)
    for u in range(NU):
        nr = jnp.max(n_e[u * 32:u * 32 + 8, :])
        ns = jnp.max(n_e[u * 32 + 16:u * 32 + 24, :])
        cnts[u] = nr
        cnts[NU + u] = ns
        cnts[2 * NU + u] = base
        base = base + ((nr + ns + 15 + (T - 1)) // T) * T

    def relayout(h):
        for c in range(8):
            rows = h * 1024 + c * 128
            xt[pl.ds(rows * 4, 512), :] = xv[pl.ds(rows, 128), :].reshape(512, 128)

    def router(r):
        _move_rows(xt, xo, ots, r * 128, r * 512, 8)
        rwb = rwv[...].astype(jnp.bfloat16)
        ei = _iota((16, 128), 0)
        xb = xo[pl.ds(r * 512, 512), :].reshape(128, D).astype(jnp.bfloat16)
        s = lax.dot_general(rwb, xb, (((1,), (1,)), ((), ())), preferred_element_type=jnp.float32)
        p = jnp.exp(s - jnp.max(s, axis=0, keepdims=True))
        probs = p / jnp.sum(p, axis=0, keepdims=True)
        a0 = jnp.sum(jnp.where(ei == oev[r:r + 1, :], probs, 0.0), axis=0, keepdims=True)
        a1 = jnp.sum(jnp.where(ei == oev[8 + r:9 + r, :], probs, 0.0), axis=0, keepdims=True)
        gs = a0 + a1
        wt = jnp.concatenate([a0 / gs, a1 / gs, jnp.zeros((126, 128), jnp.float32)], axis=0).T
        rows = pl.ds(r * 512, 512)
        g0[rows, :] = jnp.broadcast_to(wt[:, 0:1], (128, 512)).reshape(512, 128)
        g1[rows, :] = jnp.broadcast_to(wt[:, 1:2], (128, 512)).reshape(512, 128)

    def gather_unit(u):
        nr = cnts[u]
        ns = cnts[NU + u]
        b4 = cnts[2 * NU + u] * 4
        _move_rows(xt, xs, lts, u * 2 * SEG, b4, (nr + 15) >> 4)
        _move_rows(xt, xs, lts, (u * 2 + 1) * SEG, b4 + nr * 4, (ns + 15) >> 4)

    x_copy(0).wait()
    relayout(0)
    for c in eager:
        c.wait()
    for s in range(NSEG):
        @pl.when(cnts[(s >> 1) + NU * (s & 1)] > EAGER)
        def _(s=s):
            sl = pl.ds(s * SEG + EAGER, SEG - EAGER)
            c1 = pltpu.make_async_copy(ltv.at[sl], lts.at[sl], sm_sems.at[2])
            c2 = pltpu.make_async_copy(lvv.at[sl], lvs.at[sl], sm_sems.at[3])
            c1.start()
            c2.start()
            c1.wait()
            c2.wait()
    c_rw.wait()

    def gather_e(e, carry):
        gather_unit(2 * e)
        return carry
    lax.fori_loop(0, EL, gather_e, 0)
    pl.semaphore_wait(bar, 3)

    def rs_copy(src4, v):
        return pltpu.make_async_remote_copy(
            _row(pbuf, src4), _row(rbuf, v & 4092), rs_send, rs_recv.at[v >> 12],
            device_id=v & 3, device_id_type=LOGICAL)

    def self_copy(src4, v):
        return pltpu.make_async_copy(_row(pbuf, src4), _row(rbuf, v & 4092), rs_recv.at[v >> 12])

    def chunk(o, j, part=None):
        sz = CAPS[j] * 4 if part is None else CAPS[j] * 2
        lo = 0 if part is None else part * sz
        return ag.at[pl.ds(pl.multiple_of((o * (N // NCHIP) + PB[j]) * 4 + lo, 8), sz), :]

    def rc(ref, k, dev):
        return pltpu.make_async_remote_copy(ref, ref, ag_send, ag_recv.at[k],
                                            device_id=dev, device_id_type=LOGICAL)

    def self_rows(j):
        h = TR0[j] // 8
        last_in_half = j + 1 == NST or TR0[j + 1] // 8 != h

        def per_expert(e, carry):
            u = 2 * e + h
            lo = poss[4096 + (e * 16 + j) * 128]
            hi = cnts[NU + u] if last_in_half else poss[4096 + (e * 16 + j + 1) * 128]
            ls = (u * 2 + 1) * SEG + lo
            s4 = (cnts[2 * NU + u] + cnts[u] + lo) * 4
            cnt = hi - lo

            def sgrp(g, c2):
                vs = [lvs[ls + g * 4 + k] for k in range(4)]
                for k in range(4):
                    self_copy(s4 + g * 16 + k * 4, vs[k]).start()
                return c2
            lax.fori_loop(0, cnt >> 2, sgrp, 0)

            def sone(k, c2):
                self_copy(s4 + k * 4, lvs[ls + k]).start()
                return c2
            lax.fori_loop((cnt >> 2) << 2, cnt, sone, 0)
            return carry
        lax.fori_loop(0, EL, per_expert, 0)

    def summ(j):
        ch = CAPS[j] * 4
        r0 = PB[j] * 8
        self_rows(j)
        blk = rbuf.at[pl.ds(r0, 2 * ch), :]
        pltpu.make_async_copy(blk, blk, rs_recv.at[j]).wait()
        ga = g0[PB[j] * 4:PB[j] * 4 + ch, :]
        gb = g1[PB[j] * 4:PB[j] * 4 + ch, :]
        dst = pl.multiple_of((me * (N // NCHIP) + PB[j]) * 4, 8)
        l0, h0 = _unpack(rbuf[pl.ds(r0, ch), :])
        l1, h1 = _unpack(rbuf[pl.ds(r0 + ch, ch), :])
        ag[pl.ds(dst, ch), :] = _pack(ga * l0 + gb * l1, ga * h0 + gb * h1)
        rc(chunk(me, j), 4 * j + 0, right).start()
        rc(chunk(me, j), 4 * j + 1, left).start()

    def wait_own(j):
        rc(chunk(left, j), 4 * j + 0, right).wait_recv()
        rc(chunk(right, j), 4 * j + 1, left).wait_recv()

    def fwd(j):
        rc(chunk(left, j, 0), 4 * j + 2, right).start()
        rc(chunk(right, j, 1), 4 * j + 3, left).start()

    def sent(j):
        rc(chunk(me, j), 4 * j + 0, right).wait_send()
        rc(chunk(me, j), 4 * j + 1, left).wait_send()
        rc(chunk(left, j, 0), 4 * j + 2, right).wait_send()
        rc(chunk(right, j, 1), 4 * j + 3, left).wait_send()

    def finish(j):
        ntok = STAGE_ROWS[j] * 128
        rc(chunk(diag, j, 0), 4 * j + 2, right).wait_recv()
        rc(chunk(diag, j, 1), 4 * j + 3, left).wait_recv()
        for hh in range(STAGE_ROWS[j]):
            _move_rows_std(ag, fbuf, poss, 2 * (TR0[j] + hh) * 128, hh * 128, 8)
        lo, hi = _unpack(fbuf[0:ntok, :])
        out_ref[TR0[j] * 128:TR0[j] * 128 + ntok, 0:512] = lo
        out_ref[TR0[j] * 128:TR0[j] * 128 + ntok, 512:1024] = hi

    def unit(u, carry):
        e = u >> 1
        nr = cnts[u]
        ns = cnts[NU + u]
        n = nr + ns
        base = cnts[2 * NU + u]

        @pl.when(u == 1)
        def _():
            router(0)
            x_copy(1).wait()
            relayout(1)

        @pl.when((u & 1) == 1)
        def _():
            gather_unit(u)

        @pl.when((u & 1) == 0)
        def _():
            w_copy(e).wait()

        def tile(t, c):
            p0 = t * T
            off4 = pl.multiple_of((base + p0) * 4, 64)
            a = xs[pl.ds(off4, T * 4), :].reshape(T, D).astype(jnp.bfloat16)
            y = jnp.dot(a, wv[e].astype(jnp.bfloat16), preferred_element_type=jnp.float32)
            pbuf[pl.ds(off4, T * 4), :] = _pack(y[:, :512], y[:, 512:]).reshape(T * 4, 128)
            nrem = jnp.clip(nr - p0, 0, T)
            lr = u * 2 * SEG + p0

            def grp(g, c2):
                vs = [lvs[lr + g * 8 + k] for k in range(8)]
                for k in range(8):
                    rs_copy(off4 + g * 32 + k * 4, vs[k]).start()
                return c2
            lax.fori_loop(0, nrem >> 3, grp, 0)

            def one(k, c2):
                rs_copy(off4 + k * 4, lvs[lr + k]).start()
                return c2
            lax.fori_loop((nrem >> 3) << 3, nrem, one, 0)
            return c
        lax.fori_loop(0, (n + (T - 1)) // T, tile, 0)
        return carry
    lax.fori_loop(0, NU, unit, 0)

    c_pos.wait()
    summ(0)
    summ(1)
    next_router = 1
    for j in range(NST):
        if j + 2 < NST:
            summ(j + 2)
        if j + 3 < NST and PB[j + 3] + CAPS[j + 3] > 128 * next_router:
            router(next_router)
            next_router += 1
        if j == 3:
            ntot = jnp.int32(0)
            for u in range(NU):
                ntot = ntot + cnts[u]

            def ws(k, c):
                rs_copy(0, 0).wait_send()
                return c
            lax.fori_loop(0, ntot, ws, 0)
        if j >= 2:
            sent(j - 2)
        wait_own(j)
        fwd(j)
        if 0 < j < NST - 2:
            finish(j - 1)
    finish(NST - 3)
    finish(NST - 2)
    finish(NST - 1)

    sent(NST - 2)
    sent(NST - 1)


def pallas_dist_moe_top2_ep_n2048_d512_e4_h1024_kernel(x, router_W, route_idx, expert_W):
    rwt = router_W.T
    ri = route_idx.astype(jnp.int32).T.reshape(2, 16, 128).transpose(1, 0, 2).reshape(32, 128)
    i32, f32 = jnp.int32, jnp.float32
    vm, sm = pltpu.VMEM, pltpu.SMEM
    dma = pltpu.SemaphoreType.DMA
    scratch = [
        vm((N, D), f32),
        vm((N * 4, 128), f32),
        vm((EL, D, H), f32),
        vm((32, 128), i32),
        vm((16, D), f32),
        vm((NSEG * SEG,), i32),
        vm((NSEG * SEG,), i32),
        vm((96 * 128,), i32),
        vm((8 * 128,), i32),
        vm((16, 128), i32),
        sm((NSEG * SEG,), i32),
        sm((NSEG * SEG,), i32),
        sm((96 * 128,), i32),
        sm((8 * 128,), i32),
        sm((32,), i32),
        vm((XS_ROWS * 4, 128), f32),
        vm((XS_ROWS * 4, 128), i32),
        vm((1024 * 4, 128), i32),
        vm((N * 4, 128), i32),
        vm((256, 512), i32),
        vm((512 * 4, 128), f32),
        vm((512 * 4, 128), f32),
        vm((512 * 4, 128), f32),
        dma((4,)), dma((EL,)), dma((4,)), dma, dma((NST,)), dma, dma((4 * NST,)),
    ]
    return pl.pallas_call(
        _kernel,
        out_shape=pltpu.VMEM((N, H), f32),
        in_specs=[pl.BlockSpec(memory_space=pl.ANY)] * 4,
        out_specs=pl.BlockSpec(memory_space=pltpu.VMEM),
        scratch_shapes=scratch,
        compiler_params=pltpu.CompilerParams(collective_id=0, vmem_limit_bytes=100 * 1024 * 1024,
                                             disable_bounds_checks=True, disable_semaphore_checks=True),
    )(x, rwt, ri, expert_W)
```

```python
import jax
import jax.numpy as jnp
from jax import lax
from jax.experimental import pallas as pl
from jax.experimental.pallas import tpu as pltpu

N = 2048
D = 512
H = 1024
NCHIP = 4
EL = 4
STAGE_ROWS = (1, 1, 2, 2, 2, 2, 2, 2, 1, 1)
NST = len(STAGE_ROWS)
TR0 = tuple(sum(STAGE_ROWS[:j]) for j in range(NST))
CAPS = tuple(32 * r for r in STAGE_ROWS)
PB = tuple(32 * t for t in TR0)
T = 160
TS = 32
NU = 2 * EL
XS_ROWS = 4096 + NU * (T + 16)
SEG = 2048
NSEG = 2 * NU
EAGER = 256
LOGICAL = pl.DeviceIdType.LOGICAL


def _iota(shape, d):
    return lax.broadcasted_iota(jnp.int32, shape, d)


def _mm(a, b):
    return jnp.dot(a.astype(jnp.bfloat16), b.astype(jnp.bfloat16),
                   preferred_element_type=jnp.float32)


def _f(m):
    return jnp.where(m, 1.0, 0.0)


def _by_stage(trow, table):
    out = jnp.full(trow.shape, table[0], jnp.int32)
    for j in range(1, NST):
        if table[j] != table[j - 1]:
            out = out + jnp.where(trow >= TR0[j], table[j] - table[j - 1], 0)
    return out


def _compress(word, nbits, rows):
    lane = _iota(word.shape, 1)
    for b in range(nbits):
        s = 1 << b
        if s < 128:
            y = pltpu.roll(word, 128 - s, 1)
            y = jnp.where(lane < 128 - s, y, pltpu.roll(y, rows - 1, 0))
        else:
            y = pltpu.roll(word, rows - s // 128, 0)
        word = jnp.where((y & s) != 0, y, jnp.where((word & s) != 0, 0, word))
    return word


def _index_compute(ri, me):
    row = _iota((32, 128), 0)
    lane = _iota((32, 128), 1)
    par = row & 1
    even = par == 0
    chip = ri >> 2
    le = ri & 3
    e0 = jnp.where(even, ri, pltpu.roll(ri, 1, 0))
    e1 = jnp.where(even, pltpu.roll(ri, 31, 0), ri)
    a = e0 >> 2
    b = e1 >> 2
    diff = (b - a) & 3
    isdiag = diff == 2
    later = (e0 & 3) * 2 + (lane & 1) - (e1 & 3) * 2
    pref = jnp.where((diff == 0) | (later > 0), a, b)
    other = a + b - pref
    r128 = _iota((128, 128), 0)
    c128 = _iota((128, 128), 1)
    uo = jnp.concatenate([_f(r128 < c128), jnp.ones((128, 128), jnp.float32)], axis=1)
    grp = r128 >> 5
    stages = tuple(range(NST))
    sameb = (((r128 >> 5) == (c128 >> 5))
             & (_by_stage((r128 & 31) >> 1, stages) == _by_stage((c128 & 31) >> 1, stages)))
    cap = _by_stage(row >> 1, CAPS)
    lblk = _f(sameb & (c128 < r128))
    bblk = _f(sameb)

    def tile(v, k):
        return jnp.concatenate([v] * k, axis=0)

    def sel(arr, k):
        return jnp.where(k == 0, arr[0:32], jnp.where(
            k == 1, arr[32:64], jnp.where(k == 2, arr[64:96], arr[96:128])))

    evn4 = (r128 & 1) == 0
    cap4 = tile(cap, 4)

    def ranks(key):
        pt = _mm(_f(evn4 & (tile(key, 4) == grp)), uo)
        rk = (pt[:, :128] + _mm(lblk, pt[:, 128:])).astype(jnp.int32)
        return rk, _mm(bblk, pt[:, 128:]).astype(jnp.int32)

    rk1, cnt1 = ranks(jnp.where(isdiag, -1, pref))
    rk2, cnt2 = ranks(jnp.where(isdiag, pref, -1))
    used1 = jnp.minimum(cnt1, cap4)
    keep = jnp.where(isdiag, sel(rk2 + used1, pref), sel(rk1, pref)) < cap
    free = cap4 - jnp.minimum(cnt1 + cnt2, cap4)
    second = isdiag & jnp.logical_not(keep)
    rk3, cnt3 = ranks(jnp.where(second, other, -1))
    keep2 = second & (sel(rk3 - free, other) < 0)
    free = free - jnp.minimum(cnt3, free)
    f1 = free[0:32]
    f2 = f1 + free[32:64]
    f3 = f2 + free[64:96]
    pt2 = _mm(_f(even & jnp.logical_not(keep | keep2)), uo)
    rank2 = (pt2[:, :128] + _mm(lblk[:32, :32], pt2[:, 128:])).astype(jnp.int32)
    op = ((rank2 >= f1).astype(jnp.int32) + (rank2 >= f2).astype(jnp.int32)
          + (rank2 >= f3).astype(jnp.int32))
    owner = jnp.where(keep, pref, jnp.where(keep2, other, op))
    owner = jnp.where(even, owner, pltpu.roll(owner, 1, 0))
    pt3 = _mm(_f(evn4 & (tile(owner, 4) == grp)), uo)
    q = sel((pt3[:, :128] + _mm(lblk, pt3[:, 128:])).astype(jnp.int32), owner)
    q = jnp.where(even, q, pltpu.roll(q, 1, 0))
    pb = _by_stage(row >> 1, PB)
    v = ((2 * pb + par * cap + q) * 4 + owner) | (_by_stage(row >> 1, stages) << 12)
    pos4 = (owner * (N // NCHIP) + pb + q) * 4

    def stack(v):
        return jnp.concatenate([v[0:16], v[0:16], v[16:32], v[16:32]] * EL, axis=0)

    r256 = _iota((256, 128), 0)
    c256 = _iota((256, 128), 1)
    g16 = r256 >> 4
    key = jnp.where(chip == me, le * 2 + (owner == me).astype(jnp.int32), -1)
    mem = stack(key) == (g16 >> 2) * 2 + (g16 & 1)
    pe = _mm(_f(mem), uo)
    rr = _iota((256, 256), 0)
    cc = _iota((256, 256), 1)
    sameg = (rr >> 4) == (cc >> 4)
    rank_e = (pe[:, :128] + _mm(_f(sameg & (cc < rr)), pe[:, 128:])).astype(jnp.int32)
    n_e = _mm(_f(sameg), pe[:, 128:]).astype(jnp.int32)
    flat16 = (r256 & 15) * 128 + c256
    word = jnp.where(mem, (flat16 - rank_e) | (stack(v) << 11), 0)
    word = _compress(word, 11, 256)
    valid = flat16 < n_e
    orig = flat16 + (word & 2047)
    tok = (((g16 >> 1) & 1) * 8 + (orig >> 8)) * 128 + (orig & 127)
    lt = jnp.where(valid, tok * 4, 0)
    lv = jnp.where(valid, word >> 11, 0)

    ro = _iota((64, 256), 0)
    co = _iota((64, 256), 1)
    jj = ro & 15
    half = jnp.zeros_like(ro)
    start = jnp.zeros_like(ro)
    for j in range(NST):
        half = jnp.where(jj == j, TR0[j] // 8, half)
        start = jnp.where(jj == j, 2 * (TR0[j] % 8), start)
    pick = ((co >> 4) == (ro >> 4) * 4 + half * 2 + 1) & ((co & 15) < start)
    offs = _mm(_f(pick), pe[:, 128:]).astype(jnp.int32)

    flat = row * 128 + lane
    mo = even & (owner == me)
    wo = jnp.where(mo, (flat - (pb + q)) | (e0 << 12) | (e1 << 16), 0)
    wo = _compress(wo, 12, 32)[:8]
    oo = flat[:8] + (wo & 4095)
    otok4 = jnp.where(row[:8] < 4, ((oo >> 8) * 128 + (oo & 127)) * 4, 0)
    return lt, lv, n_e, jnp.concatenate([pos4, offs], axis=0), otok4, (wo >> 12) & 15, (wo >> 16) & 15


def _pack(lo, hi):
    ul = lax.bitcast_convert_type(lo, jnp.int32)
    uh = lax.bitcast_convert_type(hi, jnp.int32)
    rl = ul + 0x7FFF + ((ul >> 16) & 1)
    rh = uh + 0x7FFF + ((uh >> 16) & 1)
    return lax.shift_right_logical(rl, 16) | (rh & jnp.int32(-65536))


def _unpack(u):
    lo = lax.bitcast_convert_type(u << 16, jnp.float32)
    hi = lax.bitcast_convert_type(u & jnp.int32(-65536), jnp.float32)
    return lo, hi


def _row(ref, r4):
    return ref.at[pl.ds(pl.multiple_of(r4, 4), 4), :]


def _ld(ref, r4):
    return ref[pl.ds(pl.multiple_of(r4, 4), 4), :]


def _move_rows(src, dst, lst, l0, d4, groups):
    def grp(g, c):
        l = l0 + g * 16
        d = d4 + g * 64
        vs = [lst[l + k] for k in range(16)]
        vals = [_ld(src, vs[k]) for k in range(16)]
        for k in range(16):
            dst[pl.ds(pl.multiple_of(d + k * 4, 4), 4), :] = vals[k]
        return c
    lax.fori_loop(0, groups, grp, 0)


def _move_rows_std(src, dst, lst, l0, d0, groups):
    def grp(g, c):
        l = l0 + g * 16
        vs = [lst[l + k] for k in range(16)]
        vals = jnp.concatenate([_ld(src, vs[k]) for k in range(16)], axis=0)
        dst[pl.ds(pl.multiple_of(d0 + g * 16, 16), 16), :] = vals.reshape(16, 512)
        return c
    lax.fori_loop(0, groups, grp, 0)


def _kernel(x_hbm, rw_hbm, ri_hbm, w_hbm, out_ref,
            xv, xt, wv, riv, rwv, ltv, lvv, posv, otv, oev,
            lts, lvs, poss, ots, cnts,
            xs, pbuf, rbuf, ag, fbuf, xo, g0, g1,
            ld_sems, w_sems, sm_sems, rs_send, rs_recv, ag_send, ag_recv):
    me = lax.axis_index("i")
    left = (me + 3) % NCHIP
    right = (me + 1) % NCHIP
    diag = (me + 2) % NCHIP

    c_ri = pltpu.make_async_copy(ri_hbm, riv, ld_sems.at[0])
    c_rw = pltpu.make_async_copy(rw_hbm, rwv, ld_sems.at[1])
    c_ri.start()
    c_rw.start()

    def x_copy(h):
        sl = pl.ds(pl.multiple_of(h * 1024, 1024), 1024)
        return pltpu.make_async_copy(x_hbm.at[sl], xv.at[sl], ld_sems.at[2 + h])

    def w_copy(e):
        return pltpu.make_async_copy(w_hbm.at[e], wv.at[e], w_sems.at[e])

    x_copy(0).start()

    def start_w(e, c):
        w_copy(e).start(priority=1)

        @pl.when(e == 0)
        def _():
            x_copy(1).start(priority=1)
        return c
    lax.fori_loop(0, EL, start_w, 0)

    bar = pltpu.get_barrier_semaphore()
    for k in (1, 2, 3):
        pl.semaphore_signal(bar, inc=1, device_id=(me + k) % NCHIP, device_id_type=LOGICAL)

    c_ri.wait()
    lt, lv, n_e, pos4, otok4, oe0, oe1 = _index_compute(riv[...], me)
    ltv[...] = lt.reshape(NSEG * SEG)
    lvv[...] = lv.reshape(NSEG * SEG)
    posv[...] = pos4.reshape(96 * 128)
    otv[...] = otok4.reshape(8 * 128)
    oev[0:8, :] = oe0
    oev[8:16, :] = oe1
    eager = [pltpu.make_async_copy(otv, ots, sm_sems.at[0])]
    for s in range(NSEG):
        sl = pl.ds(s * SEG, EAGER)
        eager.append(pltpu.make_async_copy(ltv.at[sl], lts.at[sl], sm_sems.at[0]))
        eager.append(pltpu.make_async_copy(lvv.at[sl], lvs.at[sl], sm_sems.at[0]))
    for c in eager:
        c.start()
    c_pos = pltpu.make_async_copy(posv, poss, sm_sems.at[1])
    c_pos.start()
    base = jnp.int32(0)
    for u in range(NU):
        nr = jnp.max(n_e[u * 32:u * 32 + 8, :])
        ns = jnp.max(n_e[u * 32 + 16:u * 32 + 24, :])
        cnts[u] = nr
        cnts[NU + u] = ns
        cnts[2 * NU + u] = base
        n = nr + ns
        nbig = (n + (T - 3 * TS - 1)) // T
        nsmall = (jnp.maximum(n - nbig * T, 0) + (TS - 1)) // TS
        cnts[3 * NU + u] = nbig
        cnts[4 * NU + u] = nsmall
        base = base + jnp.maximum(nbig * T + nsmall * TS, ((n + 30) >> 4) << 4)

    def relayout(h):
        for c in range(8):
            rows = h * 1024 + c * 128
            xt[pl.ds(rows * 4, 512), :] = xv[pl.ds(rows, 128), :].reshape(512, 128)

    def router(r):
        _move_rows(xt, xo, ots, r * 128, r * 512, 8)
        rwb = rwv[...].astype(jnp.bfloat16)
        ei = _iota((16, 128), 0)
        xb = xo[pl.ds(r * 512, 512), :].reshape(128, D).astype(jnp.bfloat16)
        s = lax.dot_general(rwb, xb, (((1,), (1,)), ((), ())), preferred_element_type=jnp.float32)
        p = jnp.exp(s - jnp.max(s, axis=0, keepdims=True))
        probs = p / jnp.sum(p, axis=0, keepdims=True)
        a0 = jnp.sum(jnp.where(ei == oev[r:r + 1, :], probs, 0.0), axis=0, keepdims=True)
        a1 = jnp.sum(jnp.where(ei == oev[8 + r:9 + r, :], probs, 0.0), axis=0, keepdims=True)
        gs = a0 + a1
        wt = jnp.concatenate([a0 / gs, a1 / gs, jnp.zeros((126, 128), jnp.float32)], axis=0).T
        rows = pl.ds(r * 512, 512)
        g0[rows, :] = jnp.broadcast_to(wt[:, 0:1], (128, 512)).reshape(512, 128)
        g1[rows, :] = jnp.broadcast_to(wt[:, 1:2], (128, 512)).reshape(512, 128)

    def gather_unit(u):
        nr = cnts[u]
        ns = cnts[NU + u]
        b4 = cnts[2 * NU + u] * 4
        _move_rows(xt, xs, lts, u * 2 * SEG, b4, (nr + 15) >> 4)
        _move_rows(xt, xs, lts, (u * 2 + 1) * SEG, b4 + nr * 4, (ns + 15) >> 4)

    x_copy(0).wait()
    relayout(0)
    for c in eager:
        c.wait()
    for s in range(NSEG):
        @pl.when(cnts[(s >> 1) + NU * (s & 1)] > EAGER)
        def _(s=s):
            sl = pl.ds(s * SEG + EAGER, SEG - EAGER)
            c1 = pltpu.make_async_copy(ltv.at[sl], lts.at[sl], sm_sems.at[2])
            c2 = pltpu.make_async_copy(lvv.at[sl], lvs.at[sl], sm_sems.at[3])
            c1.start()
            c2.start()
            c1.wait()
            c2.wait()
    c_rw.wait()

    def gather_e(e, carry):
        gather_unit(2 * e)
        return carry
    lax.fori_loop(0, EL, gather_e, 0)
    pl.semaphore_wait(bar, 3)

    def rs_copy(src4, v):
        return pltpu.make_async_remote_copy(
            _row(pbuf, src4), _row(rbuf, v & 4092), rs_send, rs_recv.at[v >> 12],
            device_id=v & 3, device_id_type=LOGICAL)

    def self_copy(src4, v):
        return pltpu.make_async_copy(_row(pbuf, src4), _row(rbuf, v & 4092), rs_recv.at[v >> 12])

    def chunk(o, j, part=None):
        sz = CAPS[j] * 4 if part is None else CAPS[j] * 2
        lo = 0 if part is None else part * sz
        return ag.at[pl.ds(pl.multiple_of((o * (N // NCHIP) + PB[j]) * 4 + lo, 8), sz), :]

    def rc(ref, k, dev):
        return pltpu.make_async_remote_copy(ref, ref, ag_send, ag_recv.at[k],
                                            device_id=dev, device_id_type=LOGICAL)

    def self_rows(j):
        h = TR0[j] // 8
        last_in_half = j + 1 == NST or TR0[j + 1] // 8 != h

        def per_expert(e, carry):
            u = 2 * e + h
            lo = poss[4096 + (e * 16 + j) * 128]
            hi = cnts[NU + u] if last_in_half else poss[4096 + (e * 16 + j + 1) * 128]
            ls = (u * 2 + 1) * SEG + lo
            s4 = (cnts[2 * NU + u] + cnts[u] + lo) * 4
            cnt = hi - lo

            def sgrp(g, c2):
                vs = [lvs[ls + g * 4 + k] for k in range(4)]
                for k in range(4):
                    self_copy(s4 + g * 16 + k * 4, vs[k]).start()
                return c2
            lax.fori_loop(0, cnt >> 2, sgrp, 0)

            def sone(k, c2):
                self_copy(s4 + k * 4, lvs[ls + k]).start()
                return c2
            lax.fori_loop((cnt >> 2) << 2, cnt, sone, 0)
            return carry
        lax.fori_loop(0, EL, per_expert, 0)

    def summ(j):
        ch = CAPS[j] * 4
        r0 = PB[j] * 8
        self_rows(j)
        blk = rbuf.at[pl.ds(r0, 2 * ch), :]
        pltpu.make_async_copy(blk, blk, rs_recv.at[j]).wait()
        ga = g0[PB[j] * 4:PB[j] * 4 + ch, :]
        gb = g1[PB[j] * 4:PB[j] * 4 + ch, :]
        dst = pl.multiple_of((me * (N // NCHIP) + PB[j]) * 4, 8)
        l0, h0 = _unpack(rbuf[pl.ds(r0, ch), :])
        l1, h1 = _unpack(rbuf[pl.ds(r0 + ch, ch), :])
        ag[pl.ds(dst, ch), :] = _pack(ga * l0 + gb * l1, ga * h0 + gb * h1)
        rc(chunk(me, j), 4 * j + 0, right).start()
        rc(chunk(me, j), 4 * j + 1, left).start()

    def wait_own(j):
        rc(chunk(left, j), 4 * j + 0, right).wait_recv()
        rc(chunk(right, j), 4 * j + 1, left).wait_recv()

    def fwd(j):
        rc(chunk(left, j, 0), 4 * j + 2, right).start()
        rc(chunk(right, j, 1), 4 * j + 3, left).start()

    def sent(j):
        rc(chunk(me, j), 4 * j + 0, right).wait_send()
        rc(chunk(me, j), 4 * j + 1, left).wait_send()
        rc(chunk(left, j, 0), 4 * j + 2, right).wait_send()
        rc(chunk(right, j, 1), 4 * j + 3, left).wait_send()

    def finish(j):
        ntok = STAGE_ROWS[j] * 128
        rc(chunk(diag, j, 0), 4 * j + 2, right).wait_recv()
        rc(chunk(diag, j, 1), 4 * j + 3, left).wait_recv()
        for hh in range(STAGE_ROWS[j]):
            _move_rows_std(ag, fbuf, poss, 2 * (TR0[j] + hh) * 128, hh * 128, 8)
        lo, hi = _unpack(fbuf[0:ntok, :])
        out_ref[TR0[j] * 128:TR0[j] * 128 + ntok, 0:512] = lo
        out_ref[TR0[j] * 128:TR0[j] * 128 + ntok, 512:1024] = hi

    def unit(u, carry):
        e = u >> 1
        nr = cnts[u]
        base = cnts[2 * NU + u]

        @pl.when(u == 1)
        def _():
            router(0)
            x_copy(1).wait()
            relayout(1)

        @pl.when((u & 1) == 1)
        def _():
            gather_unit(u)

        @pl.when((u & 1) == 0)
        def _():
            w_copy(e).wait()

        def tile(p0, size):
            off4 = pl.multiple_of((base + p0) * 4, 64)
            a = xs[pl.ds(off4, size * 4), :].reshape(size, D).astype(jnp.bfloat16)
            y = jnp.dot(a, wv[e].astype(jnp.bfloat16), preferred_element_type=jnp.float32)
            pbuf[pl.ds(off4, size * 4), :] = _pack(y[:, :512], y[:, 512:]).reshape(size * 4, 128)
            nrem = jnp.clip(nr - p0, 0, size)
            lr = u * 2 * SEG + p0

            def grp(g, c2):
                vs = [lvs[lr + g * 8 + k] for k in range(8)]
                for k in range(8):
                    rs_copy(off4 + g * 32 + k * 4, vs[k]).start()
                return c2
            lax.fori_loop(0, nrem >> 3, grp, 0)

            def one(k, c2):
                rs_copy(off4 + k * 4, lvs[lr + k]).start()
                return c2
            lax.fori_loop((nrem >> 3) << 3, nrem, one, 0)

        nbig = cnts[3 * NU + u]

        def big(t, c):
            tile(t * T, T)
            return c
        lax.fori_loop(0, nbig, big, 0)

        def small(t, c):
            tile(nbig * T + t * TS, TS)
            return c
        lax.fori_loop(0, cnts[4 * NU + u], small, 0)
        return carry
    lax.fori_loop(0, NU, unit, 0)

    c_pos.wait()
    summ(0)
    summ(1)
    next_router = 1
    for j in range(NST):
        if j + 2 < NST:
            summ(j + 2)
        if j + 3 < NST and PB[j + 3] + CAPS[j + 3] > 128 * next_router:
            router(next_router)
            next_router += 1
        if j == 3:
            ntot = jnp.int32(0)
            for u in range(NU):
                ntot = ntot + cnts[u]

            def ws(k, c):
                rs_copy(0, 0).wait_send()
                return c
            lax.fori_loop(0, ntot, ws, 0)
        if j >= 2:
            sent(j - 2)
        wait_own(j)
        fwd(j)
        if 0 < j < NST - 2:
            finish(j - 1)
    finish(NST - 3)
    finish(NST - 2)
    finish(NST - 1)

    sent(NST - 2)
    sent(NST - 1)


def pallas_dist_moe_top2_ep_n2048_d512_e4_h1024_kernel(x, router_W, route_idx, expert_W):
    rwt = router_W.T
    ri = route_idx.astype(jnp.int32).T.reshape(2, 16, 128).transpose(1, 0, 2).reshape(32, 128)
    i32, f32 = jnp.int32, jnp.float32
    vm, sm = pltpu.VMEM, pltpu.SMEM
    dma = pltpu.SemaphoreType.DMA
    scratch = [
        vm((N, D), f32),
        vm((N * 4, 128), f32),
        vm((EL, D, H), f32),
        vm((32, 128), i32),
        vm((16, D), f32),
        vm((NSEG * SEG,), i32),
        vm((NSEG * SEG,), i32),
        vm((96 * 128,), i32),
        vm((8 * 128,), i32),
        vm((16, 128), i32),
        sm((NSEG * SEG,), i32),
        sm((NSEG * SEG,), i32),
        sm((96 * 128,), i32),
        sm((8 * 128,), i32),
        sm((5 * NU,), i32),
        vm((XS_ROWS * 4, 128), f32),
        vm((XS_ROWS * 4, 128), i32),
        vm((1024 * 4, 128), i32),
        vm((N * 4, 128), i32),
        vm((256, 512), i32),
        vm((512 * 4, 128), f32),
        vm((512 * 4, 128), f32),
        vm((512 * 4, 128), f32),
        dma((4,)), dma((EL,)), dma((4,)), dma, dma((NST,)), dma, dma((4 * NST,)),
    ]
    return pl.pallas_call(
        _kernel,
        out_shape=pltpu.VMEM((N, H), f32),
        in_specs=[pl.BlockSpec(memory_space=pl.ANY)] * 4,
        out_specs=pl.BlockSpec(memory_space=pltpu.VMEM),
        scratch_shapes=scratch,
        compiler_params=pltpu.CompilerParams(collective_id=0, vmem_limit_bytes=100 * 1024 * 1024,
                                             disable_bounds_checks=True, disable_semaphore_checks=True),
    )(x, rwt, ri, expert_W)
```
